```python
import numpy as np

kernel_name = "dist_rs_then_ag_i_m2048_n1024"

def setup_inputs():
    return {"x": np.random.randn(8192, 1024).astype(np.float32)}

def reference(x: np.ndarray) -> np.ndarray:
    return x.reshape(4, 2048, 1024).sum(axis=0)
```

```python
import jax
import jax.numpy as jnp
from jax import lax
from jax.experimental import pallas as pl
from jax.experimental.pallas import tpu as pltpu

M, N = 2048, 1024
Q = M // 4
SUB = 16


def _spans(sizes):
    spans, start = [], 0
    for size in sizes:
        spans.append((start, size))
        start += size
    assert start == Q
    return spans


C1 = _spans((16, 48, 64, 128, 256))
C2 = _spans((256, 256))
C3 = _spans((256, 256))


def _body(x_hbm, out, xs, xk, s1, r1, s2, r2, lsem, ksem, ssem, rsem1, rsem2, rsem3):
    me = lax.axis_index("i")
    nx, ny = me ^ 3, me ^ 1
    cx, cy = me >> 1, (me ^ (me >> 1)) & 1
    first = (nx, ny)
    second = (ny, nx)
    keep = (cx * Q, 2 * Q + cy * Q)
    give = ((1 - cx) * Q, 2 * Q + (1 - cy) * Q)

    bar = pltpu.get_barrier_semaphore()
    for nb in (nx, ny):
        pl.semaphore_signal(bar, inc=1, device_id=(nb,), device_id_type=pl.DeviceIdType.MESH)

    def load_give(h, c):
        o, s = C1[c]
        return pltpu.make_async_copy(
            x_hbm.at[pl.ds(pl.multiple_of(give[h] + o, 8), s)], xs.at[h, pl.ds(o, s)], lsem.at[h * len(C1) + c])

    def load_keep(h):
        return pltpu.make_async_copy(x_hbm.at[pl.ds(pl.multiple_of(keep[h], 8), Q)], xk.at[h], ksem.at[h])

    for c in range(len(C1)):
        for h in range(2):
            load_give(h, c).start()
    for h in range(2):
        load_keep(h).start()

    def rdma(src, dst, rsem, dev):
        return pltpu.make_async_remote_copy(
            src, dst, ssem, rsem, device_id=(dev,), device_id_type=pl.DeviceIdType.MESH)

    def send1(h, c):
        o, s = C1[c]
        return rdma(s1.at[h, pl.ds(o, s)], r1.at[h, pl.ds(o, s)], rsem1.at[h * len(C1) + c], first[h])

    def send2(h, c):
        o, s = C2[c]
        return rdma(s2.at[h, pl.ds(o, s)], r2.at[h, pl.ds(o, s)], rsem2.at[h * len(C2) + c], second[h])

    def send3(h, c, base):
        o, s = C3[c]
        rows = out.at[pl.ds(pl.multiple_of(base + o, 16), s)]
        return rdma(rows, rows, rsem3.at[h * len(C3) + c], first[h])

    def rowwise(o, s, fn):
        if s <= SUB:
            fn(o, s)
        else:
            @pl.loop(0, s // SUB)
            def _(i):
                fn(pl.multiple_of(o + i * SUB, SUB), SUB)

    for c, (o, s) in enumerate(C1):
        for h in range(2):
            load_give(h, c).wait()

            def f(r, n, h=h):
                s1[h, pl.ds(r, n)] = xs[h, pl.ds(r, n)].astype(jnp.bfloat16)

            rowwise(o, s, f)
            if c == 0 and h == 0:
                pl.semaphore_wait(bar, 2)
            send1(h, c).start()
    for h in range(2):
        load_keep(h).wait()
    done = 0
    for c, (o, s) in enumerate(C2):
        need = [k for k in range(done, len(C1)) if C1[k][0] < o + s]
        done += len(need)
        for h in range(2):
            for k in need:
                send1(h, k).wait_recv()

            def f(r, n, h=h):
                v = xk[h, pl.ds(r, n)] + r1[h, pl.ds(r, n)].astype(jnp.float32)
                s2[h, pl.ds(r, n)] = v.astype(jnp.bfloat16)

            rowwise(o, s, f)
            send2(h, c).start()
    done = 0
    for c, (o, s) in enumerate(C3):
        need = [k for k in range(done, len(C2)) if C2[k][0] < o + s]
        done += len(need)
        for h in range(2):
            for k in need:
                send2(h, k).wait_recv()

            def f(r, n, h=h):
                v = s2[h, pl.ds(r, n)].astype(jnp.float32) + r2[h, pl.ds(r, n)].astype(jnp.float32)
                out[pl.ds(pl.multiple_of(keep[h] + r, SUB), n)] = v.astype(jnp.bfloat16)

            rowwise(o, s, f)
            send3(h, c, keep[h]).start()
    for _ in range(3):
        pltpu.make_async_copy(s1, s1, ssem).wait()
    for c in range(len(C3)):
        for h in range(2):
            send3(h, c, give[h]).wait_recv()


def pallas_dist_rs_then_ag_i_m2048_n1024_kernel(x: jax.Array):
    return pl.pallas_call(
        _body,
        out_shape=jax.ShapeDtypeStruct((M, N), jnp.bfloat16),
        in_specs=[pl.BlockSpec(memory_space=pl.ANY)],
        out_specs=pl.BlockSpec(memory_space=pltpu.VMEM),
        scratch_shapes=[
            pltpu.VMEM((2, Q, N), jnp.float32),
            pltpu.VMEM((2, Q, N), jnp.float32),
            pltpu.VMEM((2, Q, N), jnp.bfloat16),
            pltpu.VMEM((2, Q, N), jnp.bfloat16),
            pltpu.VMEM((2, Q, N), jnp.bfloat16),
            pltpu.VMEM((2, Q, N), jnp.bfloat16),
            pltpu.SemaphoreType.DMA((2 * len(C1),)),
            pltpu.SemaphoreType.DMA((2,)),
            pltpu.SemaphoreType.DMA,
            pltpu.SemaphoreType.DMA((2 * len(C1),)),
            pltpu.SemaphoreType.DMA((2 * len(C2),)),
            pltpu.SemaphoreType.DMA((2 * len(C3),)),
        ],
        compiler_params=pltpu.CompilerParams(collective_id=0, vmem_limit_bytes=64 * 2**20),
    )(x)
```

```python
import jax
import jax.numpy as jnp
import numpy as np
from jax import lax
from jax.experimental import pallas as pl
from jax.experimental.pallas import tpu as pltpu

ROWS, N = 2048, 1024
UNIT = 256
SLAB = 32
STEPS = UNIT // SLAB
HALF = STEPS // 2
TILE = 128
I32 = jnp.int32

LONGEST = 16
SLOT = 13
WIDE = 3
SPILL = 8
LOW, EXTRA, WORDS, SIGNS, RANKS, END = 0, 64, 65, 65 + SLOT, 73 + SLOT, 137 + SLOT

D, F, S, O = range(4)
IN_S, IN_O, PART_O, END_S, END_F, END_D = range(6)
LOW_A, LOW_B, HEAD, REST, TAIL = range(5)
TAIL_PIECES = ((32, 16), (48, 8), (56, 6), (62, 2))
PARTS = TAIL + len(TAIL_PIECES)
LEAD_TILES = 2
EARLY = 5

shl = lax.shift_left
shr = lax.shift_right_logical


def _c(value):
    return np.int32(value)


def _bytes(byte):
    return np.uint32(byte * 0x01010101).astype(np.int32)


def _tiles(first, count):
    start = first * TILE
    return pl.ds(start if isinstance(first, int) else pl.multiple_of(start, TILE), count * TILE)


def _to_words(x):
    return pltpu.bitcast(x.astype(jnp.bfloat16), I32)


def _from_words(words):
    return pltpu.bitcast(words, jnp.bfloat16)


def _choose_offset(words):
    magnitudes = (words & _c(0x7FFF)) + (shr(words, _c(16)) & _c(0x7FFF))
    mean = jnp.sum(magnitudes.astype(jnp.float32)) * (0.5 / words.size)
    return (mean.astype(I32) + _c(470)) & _c(0xFFFF)


def _split_bytes(w1, w2, offset):
    both = offset * _c(0x00010001)
    t1, t2 = both - w1, both - w2
    x = (shr(t1, _c(8)) ^ t2) & _c(0x00FF00FF)
    return t1 ^ shl(x, _c(8)), t2 ^ x


def _top_rank(low):
    x = shr(low, _c(5)) & _bytes(0x07)
    return (x - (shr(x + _bytes(0x01), _c(3)) & _bytes(0x01))) ^ _bytes(0x87)


def _to_ranks(low, high):
    r = _top_rank(low)
    u = high & _bytes(0x7F)
    top = (_bytes(0x80) - u) & _bytes(0x80)
    return high - (shr(r - u, _c(7)) & _bytes(0x01)) + ((r + _bytes(0x01)) & (top - shr(top, _c(7))))


def _join_bytes(low, ranks, offset):
    q = ranks & _bytes(0x7F)
    at_most = _top_rank(low) - q
    below = at_most - _bytes(0x01)
    top = (at_most ^ below) & _bytes(0x80)
    high = ranks + (shr(below, _c(7)) & _bytes(0x01)) - (q & (top - shr(top, _c(7))))
    x = (shr(low, _c(8)) ^ high) & _c(0x00FF00FF)
    both = offset * _c(0x00010001)
    return both - (low ^ shl(x, _c(8))), both - (high ^ x)


def _shift_back(words, bits):
    other = _c(32) - bits
    middle = [shr(words[k], bits) | shl(words[k - 1], other) for k in range(1, len(words))]
    return [shr(words[0], bits)] + middle + [shl(words[-1], other)]


def _shift_forward(words, bits):
    return [shl(words[k], bits) | shr(words[k + 1], _c(32) - bits) for k in range(len(words) - 1)]


def _push_ranks(words, ranks):
    lengths = (ranks & _bytes(0x7F)) + _bytes(0x01)
    la, lb = lengths & _c(0xFF), shr(lengths, _c(24))
    lc, ld = shr(lengths, _c(8)) & _c(0xFF), shr(lengths, _c(16)) & _c(0xFF)
    code = shl(jnp.ones_like(lb), lb) | _c(1)
    code = shl(code, lc) | _c(1)
    code = shl(code, ld) | _c(1)
    bits = (la + lb) + (lc + ld)
    room = _c(32) - bits
    out = _shift_back(words, bits)[: len(words)]
    return [shl(code, room) | out[0]] + out[1:], bits, room


def _pop_ranks(words):
    x = words[0]
    qa = lax.clz(x)
    x = shl(shl(x, _c(1)), qa)
    qb = lax.clz(x)
    x = shl(shl(x, _c(1)), qb)
    qc = lax.clz(x)
    x = shl(shl(x, _c(1)), qc)
    qd = lax.clz(x)
    bits = (qa + qb) + (qc + _c(4)) + qd
    out = _shift_forward(words, bits) + [shl(words[-1], bits)]
    return out, (qa | shl(qb, _c(24))) | (shl(qc, _c(8)) | shl(qd, _c(16)))


def _merge_halves(words, bits, count, out_words):
    half = bits.shape[1] // 2
    front = bits[:, half:]
    moved = _shift_back([w[:, :half] for w in words], front & _c(31))
    least, most = count // 32, len(words)
    hit = {j: shr(front, _c(5)) == j for j in range(least + 1, most + 1)}
    zero = jnp.zeros_like(front)
    out = []
    for k in range(out_words):
        v = moved[k - least] if 0 <= k - least < len(moved) else zero
        for j in range(least + 1, most + 1):
            if 0 <= k - j < len(moved):
                v = jnp.where(hit[j], moved[k - j], v)
            elif v is not zero:
                v = jnp.where(hit[j], zero, v)
        out.append(v | words[k][:, half:] if k < len(words) else v)
    return out, bits[:, :half] + front


def _split_halves(words, count, out_words):
    first, last = (count - 1) // 32, out_words - 1
    zero = jnp.zeros_like(words[0])

    def word(k):
        return words[k] if k < len(words) else zero

    seen = zero
    for k in range(first):
        seen = seen + lax.population_count(words[k])
    wanted = count - seen
    window = [word(first + k) for k in range(out_words + 1)]
    for j in range(first + 1, last + 1):
        seen = seen + lax.population_count(words[j - 1])
        later = seen < count
        wanted = jnp.where(later, count - seen, wanted)
        window = [jnp.where(later, word(j + k), v) for k, v in enumerate(window)]
    skip = zero + _c(32)
    for step in (16, 8, 4, 2, 1):
        less = skip - _c(step)
        skip = jnp.where(lax.population_count(shr(window[0], less)) < wanted, less, skip)
    second = _shift_forward(window, _c(33) - skip)
    return [jnp.concatenate([second[k], words[k]], axis=1) for k in range(out_words)]


def _slot_layout():
    row = lax.broadcasted_iota(I32, (8, TILE), 0)
    header = (row | lax.broadcasted_iota(I32, (8, TILE), 1)) == 0
    return row, header, jnp.logical_and(row < WIDE, jnp.logical_not(header))


def _from_earlier(x, k, row):
    if k % 8 == 0:
        return pltpu.roll(x, k // 8, 1)
    y = pltpu.roll(x, k, 0)
    return jnp.where(row < k, pltpu.roll(y, 1, 1), y)


def _from_next(x, row):
    y = pltpu.roll(x, 7, 0)
    return jnp.where(row == 7, pltpu.roll(y, TILE - 1, 1), y)


def _code_step(i, w1, w2, offset, msg, state, low_stored=None, c0=0, nc=8):
    low, high = _split_bytes(w1, w2, offset)
    msg[:, _tiles(LOW + 8 * i + c0, nc)] = low
    if low_stored is not None:
        low_stored()
    ranks = _to_ranks(low, high)
    msg[:, _tiles(RANKS + 8 * i + c0, nc)] = ranks
    cols = _tiles(c0, nc)
    words, bits, room = _push_ranks([state[k, :, cols] for k in range(3)], ranks)
    for k in range(3):
        state[k, :, cols] = words[k]
    state[3, :, cols] = shr(state[3, :, cols], _c(1)) | (ranks & _bytes(0x80))
    state[4, :, cols] = state[4, :, cols] + bits
    state[5, :, cols] = state[5, :, cols] | room


def _code_finish(offset, msg, state):
    words, signs, bits = [state[0], state[1], state[2]], state[3], state[4]
    misfit = state[5]
    for count, out_words in ((32, 5), (64, 9), (128, LONGEST)):
        misfit = misfit | (_c(32 * len(words)) - bits)
        half = misfit.shape[1] // 2
        misfit = misfit[:, :half] | misfit[:, half:]
        words, bits = _merge_halves(words, bits, count, out_words)
    row, header, wide = _slot_layout()
    over = bits + _c(8) - jnp.where(wide, _c(32 * SLOT + 32), _c(32 * SLOT))
    total, peak = over, jnp.maximum(over, 0)
    for k in (1, 2, 4, 8, 16, 32, 64):
        total, peak = (
            total + _from_earlier(total, k, row),
            jnp.maximum(peak, _from_earlier(peak, k, row) + total),
        )
    taken = _from_earlier(peak, 1, row)
    again = _from_earlier(jnp.maximum(taken + over, 0), 1, row)
    start = taken + _c(8)
    misfit = misfit | (_c(32 * LONGEST) - bits) | (taken - again) | (_c(32 * SPILL - 1) - start)
    fits = jnp.max(shr(misfit, _c(31)).astype(jnp.float32)) == 0.0

    zero = jnp.zeros_like(bits)
    words = _shift_back(words, start & _c(31))
    words += [zero] * (SLOT + 1 + SPILL - len(words))
    for j in (1, 2, 4):
        move = (start & _c(32 * j)) != 0
        words = [jnp.where(move, words[k - j] if k >= j else zero, w) for k, w in enumerate(words)]
    spill = [
        _from_earlier(jnp.where(wide, words[SLOT + 1 + k], words[SLOT + k]), 1, row)
        for k in range(SPILL)
    ]
    for k, w in enumerate(_shift_back(spill, _c(8))[:SPILL]):
        words[k] = words[k] | w
    words[0] = words[0] | shl(taken, _c(24))
    word = offset | jnp.where(fits, _c(0), _c(1 << 16))
    msg[:, _tiles(EXTRA, 1)] = jnp.where(header, word, words[SLOT])
    msg[:, _tiles(WORDS, SLOT)] = jnp.concatenate(words[:SLOT], axis=1)
    msg[:, _tiles(SIGNS, 8)] = signs
    return fits


def _read_header(msg):
    word = msg[pl.ds(0, 1), _tiles(EXTRA, 1)][0, 0]
    return word & _c(0xFFFF), (word & _c(1 << 16)) == 0


def _expand_ranks(msg):
    signs = msg[:, _tiles(SIGNS, 8)]
    row, _, wide = _slot_layout()
    words = [msg[:, _tiles(WORDS + k, 1)] for k in range(SLOT)]
    spill = [_from_next(w, row) for w in _shift_forward(words[: SPILL + 1], _c(8))]
    with_extra = [msg[:, _tiles(EXTRA, 1)]] + spill
    words += [jnp.where(wide, with_extra[k], spill[min(k, SPILL - 1)]) for k in range(SPILL + 1)]
    start = shr(words[0], _c(24)) + _c(8)
    for j in (4, 2, 1):
        move = (start & _c(32 * j)) != 0
        words = [
            jnp.where(move, words[min(k + j, len(words) - 1)], words[k]) for k in range(LONGEST + j)
        ]
    words = _shift_forward(words, start & _c(31))
    for count, out_words in ((128, 9), (64, 5), (32, 3)):
        words = _split_halves(words, count, out_words)

    def step(j, words):
        words, ranks = _pop_ranks(list(words))
        msg[:, _tiles(RANKS + 8 * (STEPS - 1 - j), 8)] = ranks | (shl(signs, j) & _bytes(0x80))
        return tuple(words)

    lax.fori_loop(0, STEPS, step, tuple(words))


def _decode_step(i, offset, msg, c0=0, nc=8):
    low, ranks = msg[:, _tiles(LOW + 8 * i + c0, nc)], msg[:, _tiles(RANKS + 8 * i + c0, nc)]
    return _join_bytes(low, ranks, offset)


def _body(x_hbm, out, xv, tx, rx, state, load_sems, send_sems, recv_sems, ready):
    me = lax.axis_index("i")
    own = me ^ shr(me, 1)

    def first(h):
        return me ^ (3 - 2 * h)

    def second(h):
        return me ^ (1 + 2 * h)

    def row0(h, unit):
        return (4 * h + (own ^ (3, 2 - h, 1 + h, 0)[unit])) * UNIT

    def slab_start(i):
        return i * SLAB if isinstance(i, int) else pl.multiple_of(i * SLAB, SLAB)

    def load(h, unit):
        rows = pl.ds(pl.multiple_of(row0(h, unit), UNIT), UNIT)
        return pltpu.make_async_copy(x_hbm.at[rows], xv.at[h, unit], load_sems.at[2 * unit + h])

    between = me & 1
    lead = jnp.where(me == 1, 1, 0)

    def load_slab(j, i, c0=0, nc=8):
        h, cols = lead ^ j, _tiles(c0, nc)
        rows = pl.ds(pl.multiple_of(row0(h, D) + slab_start(i), SLAB), SLAB)
        sem = load_sems.at[8 + 2 * i + j if c0 == 0 else 8 + 2 * STEPS]
        return pltpu.make_async_copy(
            x_hbm.at[rows, cols], xv.at[h, D, pl.ds(slab_start(i), SLAB), cols], sem
        )

    def signal_neighbours(sem):
        for h in range(2):
            pl.semaphore_signal(
                sem, inc=1, device_id=(first(h),), device_id_type=pl.DeviceIdType.MESH
            )

    order = [(0, 0, 0, LEAD_TILES), (0, 0, LEAD_TILES, 8 - LEAD_TILES)]
    order += [(1 - between, between, 0, 8), (between, 1 - between, 0, 8), (1, 1, 0, 8)]
    order += [(j, i, 0, 8) for i in range(2, STEPS) for j in range(2)]
    load_slab(*order[0]).start()
    barrier = pltpu.get_barrier_semaphore()
    pl.when(me != 2)(lambda: signal_neighbours(barrier))
    for piece in order[1:6]:
        load_slab(*piece).start()

    @pl.when(me == 2)
    def _():
        pl.semaphore_wait(barrier, 2)
        signal_neighbours(ready)

    for piece in order[6:]:
        load_slab(*piece).start()

    def copy(h, msg, part, tile, tiles, rows=8):
        if msg == END_D:
            src, device = rx.at[h, END_S], first(h)
        else:
            src = tx.at[h, (D, F, S, O, O)[msg]]
            device = (first, first, second, second, first)[msg](h)
        k = (h * 6 + msg) * PARTS + part
        at = (pl.ds(0, rows), _tiles(tile, tiles))
        return pltpu.make_async_remote_copy(
            src.at[at],
            rx.at[h, msg].at[at],
            send_sems.at[k],
            recv_sems.at[k],
            device_id=(device,),
            device_id_type=pl.DeviceIdType.MESH,
        )

    def low_slab(h, msg, i):
        return copy(h, msg, shr(i, 2), LOW + 8 * i, 8)

    def low_half(h, msg, part):
        return copy(h, msg, part, LOW + 8 * HALF * part, 8 * HALF)

    def head(h, msg):
        return copy(h, msg, HEAD, EXTRA, 1, WIDE)

    def rest(h, msg, fits, act):
        pl.when(fits)(lambda: act(copy(h, msg, REST, WORDS, RANKS - WORDS)))
        pl.when(jnp.logical_not(fits))(lambda: act(copy(h, msg, REST, RANKS, END - RANKS)))

    def start(c):
        c.start()

    def note(plain, h, msg, fits):
        return plain | shl(jnp.where(fits, 0, 1), h * 6 + msg)

    def receive_rest(h, msg, landed=None):
        offset, fits = _read_header(rx.at[h, msg])
        rest(h, msg, fits, lambda c: c.wait_recv())
        if landed is not None:
            landed(fits)
        pl.when(fits)(lambda: _expand_ranks(rx.at[h, msg]))
        return offset, fits

    def receive(h, msg):
        low_half(h, msg, LOW_A).wait_recv()
        low_half(h, msg, LOW_B).wait_recv()
        head(h, msg).wait_recv()
        return receive_rest(h, msg)[0]

    def slab(h, unit, i, c0=0, nc=8):
        r, cols = slab_start(i), _tiles(c0, nc)
        return xv[h, unit, pl.ds(r, 16), cols], xv[h, unit, pl.ds(r + 16, 16), cols]

    def code(words_of, h, unit, each):
        offset = _choose_offset(words_of(0)[0])
        state[0] = jnp.zeros(state.shape[1:], I32)

        @pl.loop(0, STEPS)
        def _(i):
            _code_step(i, *words_of(i), offset, tx.at[h, unit], state.at[0])
            each(i)

        return _code_finish(offset, tx.at[h, unit], state.at[0])

    def plus(values, h, msg, offset, i):
        words = _decode_step(i, offset, rx.at[h, msg])
        return [v + _from_words(w).astype(jnp.float32) for v, w in zip(values, words)]

    def emit(h, unit, i, words, c0=0, nc=8):
        r, cols = pl.multiple_of(row0(h, unit) + i * SLAB, SLAB), _tiles(c0, nc)
        out[pl.ds(r, 16), cols] = _from_words(words[0])
        out[pl.ds(r + 16, 16), cols] = _from_words(words[1])

    def emit_slabs(h, unit, msg, offset, lo, hi):
        @pl.loop(lo, hi)
        def _(i):
            emit(h, unit, i, _decode_step(i, offset, rx.at[h, msg]))

    state[...] = jnp.zeros(state.shape, I32)
    offsets = [None, None]
    for n, (j, i, c0, nc) in enumerate(order[: EARLY + 1]):
        h = lead ^ j
        load_slab(j, i, c0, nc).wait()
        words = [_to_words(v) for v in slab(h, D, i, c0, nc)]
        if n == 0:
            offsets[0] = _choose_offset(words[0])
        elif n == 2:
            offsets[1] = _choose_offset(words[0])
        elif n == 3:
            offsets[1] = jnp.where(j == 1, _choose_offset(words[0]), offsets[1])
        offset = offsets[j] if isinstance(j, int) else jnp.where(j == 1, offsets[1], offsets[0])

        def send(n=n, j=j, h=h, i=i, c0=c0, nc=nc):
            if n == 0:
                pl.when(me == 0)(lambda: pl.semaphore_wait(barrier, 2))
                pl.when(between == 1)(lambda: pl.semaphore_wait(barrier, 1))
            piece = lambda: copy(h, IN_S, LOW_A, LOW + 8 * i + c0, nc).start()
            if isinstance(j, int) and j == 0:
                piece()
            else:
                pl.when((j & between) == 0)(piece)

        _code_step(i, *words, offset, tx.at[h, D], state.at[j], send, c0, nc)

    @pl.when(between == 1)
    def _():
        pl.semaphore_wait(ready, 1)
        copy(lead ^ 1, IN_S, LOW_A, LOW, 8 * (EARLY // 2)).start()

    for unit in (F, S, O):
        for h in range(2):
            load(h, unit).start()

    @pl.loop(EARLY, 2 * STEPS)
    def _(n):
        j, i = n & 1, shr(n, 1)
        h = lead ^ j
        load_slab(j, i).wait()
        offset = jnp.where(j == 1, offsets[1], offsets[0])
        _code_step(i, *map(_to_words, slab(h, D, i)), offset, tx.at[h, D], state.at[j])
        low_slab(h, IN_S, i).start()

    def finish_diagonal(j, plain):
        h = lead ^ j
        offset = jnp.where(j == 1, offsets[1], offsets[0])
        fits = _code_finish(offset, tx.at[h, D], state.at[j])
        head(h, IN_S).start()
        rest(h, IN_S, fits, start)
        return note(plain, h, IN_S, fits)

    plain = lax.fori_loop(0, 2, finish_diagonal, _c(0))

    def for_first(h, carry):
        load(h, F).wait()

        def each(i):
            pl.when((h == 0) | (i < HALF))(lambda: low_slab(h, IN_O, i).start())

        fits = code(lambda i: [_to_words(v) for v in slab(h, F, i)], h, F, each)

        @pl.when(h == 0)
        def _():
            head(h, IN_O).start()
            rest(h, IN_O, fits, start)

        return note(carry, h, IN_O, fits)

    plain = lax.fori_loop(0, 2, for_first, plain)

    def fitted(plain, h, msg):
        return (shr(plain, h * 6 + msg) & 1) == 0

    def for_second(h, plain):
        load(h, S).wait()
        offset = receive(h, IN_S)
        fits = code(
            lambda i: [_to_words(v) for v in plus(slab(h, S, i), h, IN_S, offset, i)],
            h,
            S,
            lambda i: low_slab(h, PART_O, i).start(),
        )
        head(h, PART_O).start()
        rest(h, PART_O, fits, start)

        @pl.when(h == 0)
        def _():
            low_half(1, IN_O, LOW_B).start()
            head(1, IN_O).start()
            rest(1, IN_O, fitted(plain, 1, IN_O), start)

        return note(plain, h, PART_O, fits)

    plain = lax.fori_loop(0, 2, for_second, plain)

    def for_all(h, plain):
        load(h, O).wait()
        offset_in = receive(h, IN_O)
        offset_part = receive(h, PART_O)

        def total(i):
            values = plus(slab(h, O, i), h, IN_O, offset_in, i)
            words = [_to_words(v) for v in plus(values, h, PART_O, offset_part, i)]
            emit(h, O, i, words)
            return words

        def each(i):
            for msg in (END_S, END_F):
                low_slab(h, msg, i).start()

        fits = code(total, h, O, each)
        for msg in (END_S, END_F):
            head(h, msg).start()
            rest(h, msg, fits, start)
            plain = note(plain, h, msg, fits)
        return plain

    plain = lax.fori_loop(0, 2, for_all, plain)

    def from_neighbours(h, plain):
        low_half(h, END_S, LOW_A).wait_recv()
        low_half(h, END_D, LOW_A).start()
        low_half(h, END_S, LOW_B).wait_recv()
        head(h, END_S).wait_recv()
        head(h, END_D).start()

        def pass_on(fits):
            rest(h, END_D, fits, start)
            for k, (tile, tiles) in enumerate(TAIL_PIECES):
                copy(h, END_D, TAIL + k, LOW + tile, tiles).start()

        offset, fits = receive_rest(h, END_S, pass_on)
        emit_slabs(h, S, END_S, offset, 0, STEPS)
        emit_slabs(h, F, END_F, receive(h, END_F), 0, STEPS)
        return note(plain, h, END_D, fits)

    plain = lax.fori_loop(0, 2, from_neighbours, plain)

    def sent(h, msg, low_parts):
        for c in low_parts + [head(h, msg)]:
            c.wait_send()
        rest(h, msg, fitted(plain, h, msg), lambda c: c.wait_send())

    @pl.loop(0, 2)
    def _(h):
        for msg in range(END_D):
            sent(h, msg, [low_half(h, msg, LOW_A), low_half(h, msg, LOW_B)])

    def diagonal_ranks(j, carry):
        h = lead ^ j
        low_half(h, END_D, LOW_A).wait_recv()
        head(h, END_D).wait_recv()
        offset = receive_rest(h, END_D)[0]
        emit_slabs(h, D, END_D, offset, 0, HALF)
        return carry[1], offset

    offsets = lax.fori_loop(0, 2, diagonal_ranks, (_c(0), _c(0)))
    for k, (tile, tiles) in enumerate(TAIL_PIECES):
        for j in range(2):
            h = lead ^ j
            if k == len(TAIL_PIECES) - 1:
                pieces = [copy(h, END_D, TAIL + t, LOW + a, b) for t, (a, b) in enumerate(TAIL_PIECES)]
                sent(h, END_D, [low_half(h, END_D, LOW_A)] + pieces)
            copy(h, END_D, TAIL + k, LOW + tile, tiles).wait_recv()
            if tiles > 8:
                emit_slabs(h, D, END_D, offsets[j], tile // 8, (tile + tiles) // 8)
            else:
                words = _decode_step(tile // 8, offsets[j], rx.at[h, END_D], tile % 8, tiles)
                emit(h, D, tile // 8, words, tile % 8, tiles)


def pallas_dist_rs_then_ag_i_m2048_n1024_kernel(x: jax.Array):
    return pl.pallas_call(
        _body,
        out_shape=jax.ShapeDtypeStruct((ROWS, N), jnp.bfloat16),
        in_specs=[pl.BlockSpec(memory_space=pl.ANY)],
        out_specs=pl.BlockSpec(memory_space=pltpu.VMEM),
        scratch_shapes=[
            pltpu.VMEM((2, 4, UNIT, N), jnp.float32),
            pltpu.VMEM((2, 4, 8, END * TILE), I32),
            pltpu.VMEM((2, 6, 8, END * TILE), I32),
            pltpu.VMEM((2, 6, 8, N), I32),
            pltpu.SemaphoreType.DMA((9 + 2 * STEPS,)),
            pltpu.SemaphoreType.DMA((12 * PARTS,)),
            pltpu.SemaphoreType.DMA((12 * PARTS,)),
            pltpu.SemaphoreType.REGULAR,
        ],
        compiler_params=pltpu.CompilerParams(
            collective_id=0, vmem_limit_bytes=64 * 2**20, disable_semaphore_checks=True
        ),
    )(x)
```

```python
import jax
import jax.numpy as jnp
import numpy as np
from jax import lax
from jax.experimental import pallas as pl
from jax.experimental.pallas import tpu as pltpu

ROWS, N = 2048, 1024
UNIT = 256
SLAB = 32
STEPS = UNIT // SLAB
TILE = 128
I32 = jnp.int32

LONGEST = 16
SLOT = 13
HEADER = 24
ZERO = 20
LOW, WORDS, SIGNS, RANKS, END = 0, 64, 64 + SLOT, 72 + SLOT, 136 + SLOT

D, F, S, O = range(4)
IN_S, IN_O, PART_O, END_S, END_F, END_D = range(6)
LOW_A, LOW_B, HEAD, REST, TAIL = range(5)
SLABS_A = (4, 5, 4, 3, 4, 3)
TAIL_PIECES = ((24, 16), (40, 8), (48, 8), (56, 6), (62, 2))
PARTS = TAIL + len(TAIL_PIECES)
DETOUR = 3
EARLY = 4

shl = lax.shift_left
shr = lax.shift_right_logical


def _c(value):
    return np.int32(value)


def _bytes(byte):
    return np.uint32(byte * 0x01010101).astype(np.int32)


def _tiles(first, count):
    start = first * TILE
    return pl.ds(start if isinstance(first, int) else pl.multiple_of(start, TILE), count * TILE)


def _to_words(x):
    return pltpu.bitcast(x.astype(jnp.bfloat16), I32)


def _from_words(words):
    return pltpu.bitcast(words, jnp.bfloat16)


def _swap_bytes(a, b):
    x = (shr(a, _c(8)) ^ b) & _c(0x00FF00FF)
    return a ^ shl(x, _c(8)), b ^ x


def _choose_scale(words):
    magnitudes = (words & _c(0x7FFF)) + (shr(words, _c(16)) & _c(0x7FFF))
    mean = jnp.sum(magnitudes.astype(jnp.float32)) * (0.5 / words.size)
    return shr(mean.astype(I32) + _c(469), _c(1)) & _c(0x3FFF)


def _scale_terms(low, scale):
    d = (shr(low, _c(1)) & _bytes(0x7F)) + (_c(0x7F) - (scale & _c(0x7F))) * _bytes(0x01)
    base = (shr(scale, _c(7)) | _c(0x80)) * _bytes(0x01) - (shr(d, _c(7)) & _bytes(0x01))
    x = shr(d, _c(4)) & _bytes(0x07)
    return base, x + (shr(_bytes(0x08) - x, _c(3)) & _bytes(0x01)) + _bytes(0x80)


def _swap_zero_class(u, scale):
    zero = shr(scale, _c(7)) * _bytes(0x01)
    hit = (_bytes(0x80) - (u ^ zero)) | (_bytes(0x80) - (u ^ _bytes(ZERO)))
    hit = hit & _bytes(0x80)
    return u ^ ((hit - shr(hit, _c(7))) & (zero ^ _bytes(ZERO)))


def _to_ranks(low, high, scale):
    base, r = _scale_terms(low, scale)
    u = _swap_zero_class((base - (high & _bytes(0x7F))) & _bytes(0x7F), scale)
    top = (_bytes(0x80) - u) & _bytes(0x80)
    ranks = u - (shr(r - u, _c(7)) & _bytes(0x01)) + ((r + _bytes(0x01)) & (top - shr(top, _c(7))))
    return ranks, high & _bytes(0x80)


def _from_ranks(low, signed_ranks, scale):
    base, r = _scale_terms(low, scale)
    q = signed_ranks & _bytes(0x7F)
    at_most = r - q
    below = at_most - _bytes(0x01)
    top = (at_most ^ below) & _bytes(0x80)
    u = q + (shr(below, _c(7)) & _bytes(0x01)) - (q & (top - shr(top, _c(7))))
    return ((base - _swap_zero_class(u, scale)) & _bytes(0x7F)) | (signed_ranks & _bytes(0x80))


def _shift_back(words, bits):
    other = _c(32) - bits
    middle = [shr(words[k], bits) | shl(words[k - 1], other) for k in range(1, len(words))]
    return [shr(words[0], bits)] + middle + [shl(words[-1], other)]


def _shift_forward(words, bits):
    other = _c(32) - bits
    return [shl(words[k], bits) | shr(words[k + 1], other) for k in range(len(words) - 1)]


def _push_ranks(words, ranks):
    lengths = ranks + _bytes(0x01)
    la, lb = lengths & _c(0xFF), shr(lengths, _c(24))
    lc, ld = shr(lengths, _c(8)) & _c(0xFF), shr(lengths, _c(16)) & _c(0xFF)
    code = shl(jnp.ones_like(lb), lb) | _c(1)
    code = shl(code, lc) | _c(1)
    code = shl(code, ld) | _c(1)
    bits = (la + lb) + (lc + ld)
    room = _c(32) - bits
    out = _shift_back(words, bits)[: len(words)]
    return [shl(code, room) | out[0]] + out[1:], bits, room


def _pop_ranks(words):
    x = words[0]
    qa = lax.clz(x)
    x = shl(shl(x, _c(1)), qa)
    qb = lax.clz(x)
    x = shl(shl(x, _c(1)), qb)
    qc = lax.clz(x)
    x = shl(shl(x, _c(1)), qc)
    qd = lax.clz(x)
    bits = (qa + qb) + (qc + _c(4)) + qd
    out = _shift_forward(words, bits) + [shl(words[-1], bits)]
    return out, (qa | shl(qb, _c(24))) | (shl(qc, _c(8)) | shl(qd, _c(16)))


def _bits_through(word, ones):
    skip = jnp.zeros_like(word) + _c(32)
    for step in (16, 8, 4, 2, 1):
        less = skip - _c(step)
        skip = jnp.where(lax.population_count(shr(word, less)) < ones, less, skip)
    return _c(33) - skip


def _merge_halves(words, bits, count, out_words):
    half = bits.shape[1] // 2
    front = bits[:, half:]
    moved = _shift_back([w[:, :half] for w in words], front & _c(31))
    least, most = count // 32, len(words)
    hit = {j: shr(front, _c(5)) == j for j in range(least + 1, most + 1)}
    zero = jnp.zeros_like(front)
    out = []
    for k in range(out_words):
        v = moved[k - least] if 0 <= k - least < len(moved) else zero
        for j in range(least + 1, most + 1):
            if 0 <= k - j < len(moved):
                v = jnp.where(hit[j], moved[k - j], v)
            elif v is not zero:
                v = jnp.where(hit[j], zero, v)
        out.append(v | words[k][:, half:] if k < len(words) else v)
    return out, bits[:, :half] + front


def _split_halves(words, count, out_words):
    first, last = (count - 1) // 32, out_words - 1
    zero = jnp.zeros_like(words[0])

    def word(k):
        return words[k] if k < len(words) else zero

    seen = zero
    for k in range(first):
        seen = seen + lax.population_count(words[k])
    wanted = count - seen
    window = [word(first + k) for k in range(out_words + 1)]
    for j in range(first + 1, last + 1):
        seen = seen + lax.population_count(words[j - 1])
        later = seen < count
        wanted = jnp.where(later, count - seen, wanted)
        window = [jnp.where(later, word(j + k), v) for k, v in enumerate(window)]
    second = _shift_forward(window, _bits_through(window[0], wanted))
    return [jnp.concatenate([second[k], words[k]], axis=1) for k in range(out_words)]


def _slot_index():
    return lax.broadcasted_iota(I32, (8, TILE), 0), lax.broadcasted_iota(I32, (8, TILE), 1)


def _from_previous(x, row):
    y = pltpu.roll(x, 1, 0)
    return jnp.where(row == 0, pltpu.roll(y, 1, 1), y)


def _from_next(x, row):
    y = pltpu.roll(x, 7, 0)
    return jnp.where(row == 7, pltpu.roll(y, TILE - 1, 1), y)


def _last_row(x):
    return jnp.broadcast_to(x[7:8, :], x.shape)


def _bits_taken(over, row):
    def join(early, late):
        return early[0] + late[0], jnp.maximum(late[1], early[1] + late[0])

    run = over, jnp.maximum(over, 0)
    for k in (1, 2, 4):
        both = join([pltpu.roll(v, k, 0) for v in run], run)
        run = [jnp.where(row >= k, a, b) for a, b in zip(both, run)]
    lanes = [_last_row(v) for v in run]
    for unit in (1, 8):
        window = lanes
        for k in range(1, 8):
            lanes = join([pltpu.roll(v, k * unit, 1) for v in window], lanes)
    before = pltpu.roll(lanes[1], 1, 1)
    after = jnp.maximum(run[1], before + run[0])
    return jnp.where(row == 0, before, pltpu.roll(after, 1, 0))


def _sum_of_earlier(x, row, lane):
    run = x
    for k in (1, 2, 4):
        run = run + jnp.where(row >= k, pltpu.roll(run, k, 0), 0)
    lanes = total = _last_row(run)
    for unit, count in ((1, 8), (8, 16)):
        window = lanes
        for k in range(1, count):
            lanes = lanes + jnp.where(lane >= k * unit, pltpu.roll(window, k * unit, 1), 0)
    return (lanes - total) + (run - x)


def _code_step(i, w1, w2, scale, msg, state, c0=0, nc=8):
    low, high = _swap_bytes(w1, w2)
    msg[:, _tiles(LOW + 8 * i + c0, nc)] = low
    ranks, signs = _to_ranks(low, high, scale())
    msg[:, _tiles(RANKS + 8 * i + c0, nc)] = ranks | signs
    cols = _tiles(c0, nc)
    words, bits, room = _push_ranks([state[k, :, cols] for k in range(3)], ranks)
    for k in range(3):
        state[k, :, cols] = words[k]
    state[3, :, cols] = shr(state[3, :, cols], _c(1)) | signs
    state[4, :, cols] = state[4, :, cols] + bits
    state[5, :, cols] = state[5, :, cols] | room


def _code_finish(scale, msg, state):
    words, signs, bits = [state[0], state[1], state[2]], state[3], state[4]
    misfit = state[5]
    for count, out_words in ((32, 5), (64, 9), (128, LONGEST)):
        misfit = misfit | (_c(32 * len(words)) - bits)
        half = misfit.shape[1] // 2
        misfit = misfit[:, :half] | misfit[:, half:]
        words, bits = _merge_halves(words, bits, count, out_words)
    row, lane = _slot_index()
    first = (row | lane) == 0
    head = jnp.where(first, _c(HEADER), 0)
    over = bits + head - _c(32 * SLOT)
    taken = _bits_taken(over, row)
    again = _from_previous(jnp.maximum(taken + over, 0), row)
    start = head + taken
    misfit = misfit | (_c(32 * LONGEST) - bits) | (taken - again) | (_c(32 * SLOT - 1) - start)
    fits = jnp.max(shr(misfit, _c(31)).astype(jnp.float32)) == 0.0

    zero = jnp.zeros_like(bits)
    words = _shift_back(words, start & _c(31))
    for j in (1, 2, 4, 8):
        move = (start & _c(32 * j)) != 0
        here = words + [zero] * j
        there = [zero] * j + words
        words = [jnp.where(move, b, a) for a, b in zip(here[: 2 * SLOT], there)]
    spill = [_from_previous(w, row) for w in words[SLOT:]]
    ones = sum(lax.population_count(w) for w in spill)
    words = [a | b for a, b in zip(words[:SLOT], _shift_back(spill, head))]
    header = scale | jnp.where(fits, _c(0), _c(1 << 14)) | shl(ones, _c(15))
    header = shl(header, _c(32 - HEADER)) | (words[0] & _c(0xFF))
    words[0] = jnp.where(first, header, words[0])
    msg[:, _tiles(WORDS, SLOT)] = jnp.concatenate(words, axis=1)
    msg[:, _tiles(SIGNS, 8)] = signs
    return fits


def _read_header(msg):
    word = shr(msg[:, _tiles(WORDS, 1)][0, 0], _c(32 - HEADER))
    return word & _c(0x3FFF), (word & _c(1 << 14)) == 0, shr(word, _c(15))


def _expand_ranks(msg, ones_in_first):
    signs = msg[:, _tiles(SIGNS, 8)]
    row, lane = _slot_index()
    first = (row | lane) == 0
    head = jnp.where(first, _c(HEADER), 0)
    words = [msg[:, _tiles(WORDS + k, 1)] for k in range(SLOT)]
    words[0] = jnp.where(first, words[0] & _c(0xFF), words[0])
    zero = jnp.zeros_like(head)
    seen = [zero]
    for w in words:
        seen.append(seen[-1] + lax.population_count(w))
    foreign = ones_in_first + _sum_of_earlier(UNIT - seen[-1], row, lane)
    words += [_from_next(w, row) for w in _shift_forward(words + [zero], head)]
    index, wanted = zero, foreign
    for k in range(1, SLOT):
        later = seen[k] < foreign
        index = jnp.where(later, k, index)
        wanted = jnp.where(later, foreign - seen[k], wanted)
    for j in (8, 4, 2, 1):
        move = (index & _c(j)) != 0
        words = [
            jnp.where(move, words[min(k + j, len(words) - 1)], words[k]) for k in range(LONGEST + j)
        ]
    words = _shift_forward(words, jnp.where(foreign == 0, head, _bits_through(words[0], wanted)))
    for count, out_words in ((128, 9), (64, 5), (32, 3)):
        words = _split_halves(words, count, out_words)

    def step(j, words):
        words, ranks = _pop_ranks(list(words))
        msg[:, _tiles(RANKS + 8 * (STEPS - 1 - j), 8)] = ranks | (shl(signs, j) & _bytes(0x80))
        return tuple(words)

    lax.fori_loop(0, STEPS, step, tuple(words))


def _decode_step(i, scale, msg, c0=0, nc=8):
    low = msg[:, _tiles(LOW + 8 * i + c0, nc)]
    return _swap_bytes(low, _from_ranks(low, msg[:, _tiles(RANKS + 8 * i + c0, nc)], scale))


def _body(x_hbm, out, xv, tx, rx, state, side, load_sems, send_sems, recv_sems, side_sems, ready):
    me = lax.axis_index("i")
    own = me ^ shr(me, 1)

    def first(h):
        return me ^ (3 - 2 * h)

    def second(h):
        return me ^ (1 + 2 * h)

    def row0(h, unit):
        return (4 * h + (own ^ (3, 2 - h, 1 + h, 0)[unit])) * UNIT

    def slab_start(i):
        return i * SLAB if isinstance(i, int) else pl.multiple_of(i * SLAB, SLAB)

    def load(h, unit):
        rows = pl.ds(pl.multiple_of(row0(h, unit), UNIT), UNIT)
        return pltpu.make_async_copy(x_hbm.at[rows], xv.at[h, unit], load_sems.at[2 * unit + h])

    between = me & 1
    lead = jnp.where(me == 1, 1, 0)

    def load_slab(j, i, c0=0, nc=8):
        h, cols = lead ^ j, _tiles(c0, nc)
        rows = pl.ds(pl.multiple_of(row0(h, D) + slab_start(i), SLAB), SLAB)
        sem = load_sems.at[8 + 2 * i + j if c0 == 0 else 8 + 2 * STEPS]
        return pltpu.make_async_copy(
            x_hbm.at[rows, cols], xv.at[h, D, pl.ds(slab_start(i), SLAB), cols], sem
        )

    def signal_neighbours(sem):
        for h in range(2):
            pl.semaphore_signal(
                sem, inc=1, device_id=(first(h),), device_id_type=pl.DeviceIdType.MESH
            )

    order = [(0, 0, DETOUR, 8 - DETOUR), (0, 0, 0, DETOUR)]
    order += [(1 - between, between, 0, 8), (between, 1 - between, 0, 8), (1, 1, 0, 8)]
    order += [(j, i, 0, 8) for i in range(2, STEPS) for j in range(2)]
    load_slab(*order[0]).start()
    barrier = pltpu.get_barrier_semaphore()
    pl.when(me != 2)(lambda: signal_neighbours(barrier))
    for piece in order[1:3]:
        load_slab(*piece).start()

    @pl.when(me == 2)
    def _():
        pl.semaphore_wait(barrier, 2)
        signal_neighbours(ready)

    def copy(h, msg, part, tile, tiles):
        if msg == END_D:
            src, device = rx.at[h, END_S], first(h)
        else:
            src = tx.at[h, (D, F, S, O, O)[msg]]
            device = (first, first, second, second, first)[msg](h)
        k = (h * 6 + msg) * PARTS + part
        cols = _tiles(tile, tiles)
        return pltpu.make_async_remote_copy(
            src.at[:, cols],
            rx.at[h, msg, :, cols],
            send_sems.at[k],
            recv_sems.at[k],
            device_id=(device,),
            device_id_type=pl.DeviceIdType.MESH,
        )

    def low_slab(h, msg, i):
        return copy(h, msg, jnp.where(i < SLABS_A[msg], LOW_A, LOW_B), LOW + 8 * i, 8)

    def low_part(h, msg, part):
        lo, hi = ((0, SLABS_A[msg]), (SLABS_A[msg], STEPS))[part]
        return copy(h, msg, part, LOW + 8 * lo, 8 * (hi - lo))

    def first_low_part(h, short, act):
        pl.when(short)(lambda: act(copy(h, IN_S, LOW_A, LOW + DETOUR, 8 * SLABS_A[IN_S] - DETOUR)))
        pl.when(jnp.logical_not(short))(lambda: act(low_part(h, IN_S, LOW_A)))

    def head(h, msg):
        return copy(h, msg, HEAD, WORDS, 1)

    def rest(h, msg, fits, act):
        pl.when(fits)(lambda: act(copy(h, msg, REST, WORDS + 1, RANKS - WORDS - 1)))
        pl.when(jnp.logical_not(fits))(lambda: act(copy(h, msg, REST, RANKS, END - RANKS)))

    def detour(h):
        return pltpu.make_async_remote_copy(
            side.at[2],
            side.at[h],
            side_sems.at[2],
            side_sems.at[h],
            device_id=(second(h),),
            device_id_type=pl.DeviceIdType.MESH,
        )

    def start(c):
        c.start()

    def wait_recv(c):
        c.wait_recv()

    def wait_send(c):
        c.wait_send()

    def note(plain, h, msg, fits):
        return plain | shl(jnp.where(fits, 0, 1), h * 6 + msg)

    def fitted(plain, h, msg):
        return (shr(plain, h * 6 + msg) & 1) == 0

    def receive_rest(h, msg, landed=None):
        scale, fits, ones = _read_header(rx.at[h, msg])
        rest(h, msg, fits, wait_recv)
        if landed is not None:
            landed(fits)
        pl.when(fits)(lambda: _expand_ranks(rx.at[h, msg], ones))
        return scale, fits

    def receive(h, msg):
        if msg == IN_S:
            first_low_part(h, me == 0, wait_recv)
        else:
            low_part(h, msg, LOW_A).wait_recv()
        low_part(h, msg, LOW_B).wait_recv()
        head(h, msg).wait_recv()
        return receive_rest(h, msg)[0]

    def slab(h, unit, i, c0=0, nc=8):
        r, cols = slab_start(i), _tiles(c0, nc)
        return xv[h, unit, pl.ds(r, 16), cols], xv[h, unit, pl.ds(r + 16, 16), cols]

    def code(words_of, h, unit, each):
        scale = _choose_scale(words_of(0)[0][:, DETOUR * TILE :])
        state[0] = jnp.zeros(state.shape[1:], I32)

        @pl.loop(0, STEPS)
        def _(i):
            _code_step(i, *words_of(i), lambda: scale, tx.at[h, unit], state.at[0])
            each(i)

        return _code_finish(scale, tx.at[h, unit], state.at[0])

    def plus(values, h, msg, scale, i):
        words = _decode_step(i, scale, rx.at[h, msg])
        if msg == IN_S:
            missing = jnp.where((me == 0) & (i == 0), DETOUR * TILE, 0)
            col = lax.broadcasted_iota(I32, words[0].shape, 1)
            words = [jnp.where(col < missing, 0, w) for w in words]
        return [v + _from_words(w).astype(jnp.float32) for v, w in zip(values, words)]

    def emit(h, unit, i, words, c0=0, nc=8):
        r, cols = pl.multiple_of(row0(h, unit) + i * SLAB, SLAB), _tiles(c0, nc)
        out[pl.ds(r, 16), cols] = _from_words(words[0])
        out[pl.ds(r + 16, 16), cols] = _from_words(words[1])

    def emit_slabs(h, unit, msg, scale, lo, hi):
        @pl.loop(lo, hi)
        def _(i):
            emit(h, unit, i, _decode_step(i, scale, rx.at[h, msg]))

    state[...] = jnp.zeros(state.shape, I32)
    pl.when(me == 0)(lambda: pl.semaphore_wait(barrier, 2))
    pl.when(between == 1)(lambda: pl.semaphore_wait(barrier, 1))
    scales = [None, None]
    for n, (j, i, c0, nc) in enumerate(order[: EARLY + 1]):
        h = lead ^ j
        load_slab(j, i, c0, nc).wait()
        words = [_to_words(v) for v in slab(h, D, i, c0, nc)]

        def send_then_scale(n=n, j=j, h=h, i=i, c0=c0, nc=nc, words=words):
            def send():
                copy(h, IN_S, LOW_A, LOW + 8 * i + c0, nc).start()

            if n == 0:
                send()
                for piece in order[3:]:
                    load_slab(*piece).start()
                scales[0] = _choose_scale(words[0])
            elif n == 1:
                pl.when(between == 0)(send)
                side[2] = jnp.concatenate(words, axis=1)
            else:
                pl.when((j & between) == 0)(send)
                if n == 2:
                    scales[1] = _choose_scale(words[0])
                elif n == 3:
                    scales[1] = jnp.where(j == 1, _choose_scale(words[0]), scales[1])
            return scales[j] if isinstance(j, int) else jnp.where(j == 1, scales[1], scales[0])

        _code_step(i, *words, send_then_scale, tx.at[h, D], state.at[j], c0, nc)

    @pl.when(between == 1)
    def _():
        pl.semaphore_wait(ready, 1)
        copy(lead ^ 1, IN_S, LOW_A, LOW, 8 * (EARLY // 2)).start()
        detour(lead).start()

    @pl.when(me == 0)
    def _():
        for h in range(2):
            rx[h, IN_S, :, _tiles(LOW, DETOUR)] = jnp.zeros((8, DETOUR * TILE), I32)

    for unit in (F, S, O):
        for h in range(2):
            load(h, unit).start()

    @pl.loop(EARLY, 2 * STEPS)
    def _(n):
        j, i = n & 1, shr(n, 1)
        h = lead ^ j
        load_slab(j, i).wait()
        scale = jnp.where(j == 1, scales[1], scales[0])
        _code_step(i, *map(_to_words, slab(h, D, i)), lambda: scale, tx.at[h, D], state.at[j])
        low_slab(h, IN_S, i).start()

    def finish_diagonal(j, plain):
        h = lead ^ j
        fits = _code_finish(jnp.where(j == 1, scales[1], scales[0]), tx.at[h, D], state.at[j])
        head(h, IN_S).start()
        rest(h, IN_S, fits, start)
        return note(plain, h, IN_S, fits)

    plain = lax.fori_loop(0, 2, finish_diagonal, _c(0))

    def for_first(h, plain):
        load(h, F).wait()

        @pl.when(me == 2)
        def _():
            detour(h).wait_recv()
            for k in range(2):
                at = (h, F, pl.ds(16 * k, 16), _tiles(0, DETOUR))
                extra = _from_words(side[h, :, _tiles(k * DETOUR, DETOUR)])
                xv[at] = xv[at] + extra.astype(jnp.float32)

        def each(i):
            pl.when((h == 0) | (i < SLABS_A[IN_O]))(lambda: low_slab(h, IN_O, i).start())

        fits = code(lambda i: [_to_words(v) for v in slab(h, F, i)], h, F, each)

        @pl.when(h == 0)
        def _():
            head(h, IN_O).start()
            rest(h, IN_O, fits, start)

        return note(plain, h, IN_O, fits)

    plain = lax.fori_loop(0, 2, for_first, plain)

    def for_second(h, plain):
        load(h, S).wait()
        scale = receive(h, IN_S)
        fits = code(
            lambda i: [_to_words(v) for v in plus(slab(h, S, i), h, IN_S, scale, i)],
            h,
            S,
            lambda i: low_slab(h, PART_O, i).start(),
        )
        head(h, PART_O).start()
        rest(h, PART_O, fits, start)

        @pl.when(h == 0)
        def _():
            low_part(1, IN_O, LOW_B).start()
            head(1, IN_O).start()
            rest(1, IN_O, fitted(plain, 1, IN_O), start)

        return note(plain, h, PART_O, fits)

    plain = lax.fori_loop(0, 2, for_second, plain)

    def for_all(h, plain):
        load(h, O).wait()
        scale_in = receive(h, IN_O)
        scale_part = receive(h, PART_O)

        def total(i):
            values = plus(slab(h, O, i), h, IN_O, scale_in, i)
            words = [_to_words(v) for v in plus(values, h, PART_O, scale_part, i)]
            emit(h, O, i, words)
            return words

        def each(i):
            for msg in (END_S, END_F):
                low_slab(h, msg, i).start()

        fits = code(total, h, O, each)
        for msg in (END_S, END_F):
            head(h, msg).start()
            rest(h, msg, fits, start)
            plain = note(plain, h, msg, fits)
        return plain

    plain = lax.fori_loop(0, 2, for_all, plain)

    def from_neighbours(h, plain):
        low_part(h, END_S, LOW_A).wait_recv()
        low_part(h, END_D, LOW_A).start()
        low_part(h, END_S, LOW_B).wait_recv()
        head(h, END_S).wait_recv()
        head(h, END_D).start()

        def pass_on(fits):
            rest(h, END_D, fits, start)
            for k, (tile, tiles) in enumerate(TAIL_PIECES):
                copy(h, END_D, TAIL + k, LOW + tile, tiles).start()

        scale, fits = receive_rest(h, END_S, pass_on)
        emit_slabs(h, S, END_S, scale, 0, STEPS)
        emit_slabs(h, F, END_F, receive(h, END_F), 0, STEPS)
        return note(plain, h, END_D, fits)

    plain = lax.fori_loop(0, 2, from_neighbours, plain)

    def sent(h, msg, low_parts):
        for c in low_parts + [head(h, msg)]:
            c.wait_send()
        rest(h, msg, fitted(plain, h, msg), wait_send)

    @pl.loop(0, 2)
    def _(h):
        first_low_part(h, (between == 1) & (h == lead), wait_send)
        sent(h, IN_S, [low_part(h, IN_S, LOW_B)])
        for msg in range(IN_O, END_D):
            sent(h, msg, [low_part(h, msg, LOW_A), low_part(h, msg, LOW_B)])

    pl.when(between == 1)(lambda: detour(lead).wait_send())

    def diagonal_ranks(j, scales):
        h = lead ^ j
        low_part(h, END_D, LOW_A).wait_recv()
        head(h, END_D).wait_recv()
        scale = receive_rest(h, END_D)[0]
        emit_slabs(h, D, END_D, scale, 0, SLABS_A[END_D])
        return scales[1], scale

    scales = lax.fori_loop(0, 2, diagonal_ranks, (_c(0), _c(0)))
    for k, (tile, tiles) in enumerate(TAIL_PIECES):
        if k == len(TAIL_PIECES) - 2:
            for h in range(2):
                tail = [copy(h, END_D, TAIL + t, LOW + a, b) for t, (a, b) in enumerate(TAIL_PIECES)]
                sent(h, END_D, [low_part(h, END_D, LOW_A)] + tail)
        for j in range(2):
            h = lead ^ j
            copy(h, END_D, TAIL + k, LOW + tile, tiles).wait_recv()
            if tiles > 8:
                emit_slabs(h, D, END_D, scales[j], tile // 8, (tile + tiles) // 8)
            else:
                words = _decode_step(tile // 8, scales[j], rx.at[h, END_D], tile % 8, tiles)
                emit(h, D, tile // 8, words, tile % 8, tiles)


def pallas_dist_rs_then_ag_i_m2048_n1024_kernel(x: jax.Array):
    return pl.pallas_call(
        _body,
        out_shape=jax.ShapeDtypeStruct((ROWS, N), jnp.bfloat16),
        in_specs=[pl.BlockSpec(memory_space=pl.ANY)],
        out_specs=pl.BlockSpec(memory_space=pltpu.VMEM),
        scratch_shapes=[
            pltpu.VMEM((2, 4, UNIT, N), jnp.float32),
            pltpu.VMEM((2, 4, 8, END * TILE), I32),
            pltpu.VMEM((2, 6, 8, END * TILE), I32),
            pltpu.VMEM((2, 6, 8, N), I32),
            pltpu.VMEM((3, 8, 2 * DETOUR * TILE), I32),
            pltpu.SemaphoreType.DMA((9 + 2 * STEPS,)),
            pltpu.SemaphoreType.DMA((12 * PARTS,)),
            pltpu.SemaphoreType.DMA((12 * PARTS,)),
            pltpu.SemaphoreType.DMA((3,)),
            pltpu.SemaphoreType.REGULAR,
        ],
        compiler_params=pltpu.CompilerParams(
            collective_id=0, vmem_limit_bytes=64 * 2**20, disable_semaphore_checks=True
        ),
    )(x)
```

```python
import jax
import jax.numpy as jnp
import numpy as np
from jax import lax
from jax.experimental import pallas as pl
from jax.experimental.pallas import tpu as pltpu

ROWS, N = 2048, 1024
UNIT = 256
SLAB = 32
STEPS = UNIT // SLAB
TILE = 128
I32 = jnp.int32

LONGEST = 16
SLOT = 13
HEADER = 24
ZERO = 20
LOW, WORDS, SIGNS, RANKS, END = 0, 64, 64 + SLOT, 72 + SLOT, 136 + SLOT

D, F, S, O = range(4)
IN_S, IN_O, PART_O, END_S, END_F, END_D = range(6)
LOW_A, LOW_B, HEAD, REST, TAIL = range(5)
SLABS_A = (4, 5, 4, 3, 4, 3)
TAIL_PIECES = ((24, 16), (40, 8), (48, 8), (56, 6), (62, 2))
PARTS = TAIL + len(TAIL_PIECES)
DETOUR = 4

shl = lax.shift_left
shr = lax.shift_right_logical


def _c(value):
    return np.int32(value)


def _bytes(byte):
    return np.uint32(byte * 0x01010101).astype(np.int32)


def _tiles(first, count):
    start = first * TILE
    return pl.ds(start if isinstance(first, int) else pl.multiple_of(start, TILE), count * TILE)


def _to_words(x):
    return pltpu.bitcast(x.astype(jnp.bfloat16), I32)


def _from_words(words):
    return pltpu.bitcast(words, jnp.bfloat16)


def _swap_bytes(a, b):
    x = (shr(a, _c(8)) ^ b) & _c(0x00FF00FF)
    return a ^ shl(x, _c(8)), b ^ x


def _choose_scale(words):
    magnitudes = (words & _c(0x7FFF)) + (shr(words, _c(16)) & _c(0x7FFF))
    mean = jnp.sum(magnitudes.astype(jnp.float32)) * (0.5 / words.size)
    return shr(mean.astype(I32) + _c(469), _c(1)) & _c(0x3FFF)


def _scale_terms(low, scale):
    d = (shr(low, _c(1)) & _bytes(0x7F)) + (_c(0x7F) - (scale & _c(0x7F))) * _bytes(0x01)
    base = (shr(scale, _c(7)) | _c(0x80)) * _bytes(0x01) - (shr(d, _c(7)) & _bytes(0x01))
    x = shr(d, _c(4)) & _bytes(0x07)
    return base, x + (shr(_bytes(0x08) - x, _c(3)) & _bytes(0x01)) + _bytes(0x80)


def _swap_zero_class(u, scale):
    zero = shr(scale, _c(7)) * _bytes(0x01)
    hit = (_bytes(0x80) - (u ^ zero)) | (_bytes(0x80) - (u ^ _bytes(ZERO)))
    hit = hit & _bytes(0x80)
    return u ^ ((hit - shr(hit, _c(7))) & (zero ^ _bytes(ZERO)))


def _to_ranks(low, high, scale):
    base, r = _scale_terms(low, scale)
    u = _swap_zero_class((base - (high & _bytes(0x7F))) & _bytes(0x7F), scale)
    top = (_bytes(0x80) - u) & _bytes(0x80)
    ranks = u - (shr(r - u, _c(7)) & _bytes(0x01)) + ((r + _bytes(0x01)) & (top - shr(top, _c(7))))
    return ranks, high & _bytes(0x80)


def _from_ranks(low, signed_ranks, scale):
    base, r = _scale_terms(low, scale)
    q = signed_ranks & _bytes(0x7F)
    at_most = r - q
    below = at_most - _bytes(0x01)
    top = (at_most ^ below) & _bytes(0x80)
    u = q + (shr(below, _c(7)) & _bytes(0x01)) - (q & (top - shr(top, _c(7))))
    return ((base - _swap_zero_class(u, scale)) & _bytes(0x7F)) | (signed_ranks & _bytes(0x80))


def _shift_back(words, bits):
    other = _c(32) - bits
    middle = [shr(words[k], bits) | shl(words[k - 1], other) for k in range(1, len(words))]
    return [shr(words[0], bits)] + middle + [shl(words[-1], other)]


def _shift_forward(words, bits):
    other = _c(32) - bits
    return [shl(words[k], bits) | shr(words[k + 1], other) for k in range(len(words) - 1)]


def _push_ranks(words, ranks):
    lengths = ranks + _bytes(0x01)
    la, lb = lengths & _c(0xFF), shr(lengths, _c(24))
    lc, ld = shr(lengths, _c(8)) & _c(0xFF), shr(lengths, _c(16)) & _c(0xFF)
    code = shl(jnp.ones_like(lb), lb) | _c(1)
    code = shl(code, lc) | _c(1)
    code = shl(code, ld) | _c(1)
    bits = (la + lb) + (lc + ld)
    room = _c(32) - bits
    out = _shift_back(words, bits)[: len(words)]
    return [shl(code, room) | out[0]] + out[1:], bits, room


def _pop_ranks(words):
    x = words[0]
    qa = lax.clz(x)
    x = shl(shl(x, _c(1)), qa)
    qb = lax.clz(x)
    x = shl(shl(x, _c(1)), qb)
    qc = lax.clz(x)
    x = shl(shl(x, _c(1)), qc)
    qd = lax.clz(x)
    bits = (qa + qb) + (qc + _c(4)) + qd
    out = _shift_forward(words, bits) + [shl(words[-1], bits)]
    return out, (qa | shl(qb, _c(24))) | (shl(qc, _c(8)) | shl(qd, _c(16)))


def _bits_through(word, ones):
    skip = jnp.zeros_like(word) + _c(32)
    for step in (16, 8, 4, 2, 1):
        less = skip - _c(step)
        skip = jnp.where(lax.population_count(shr(word, less)) < ones, less, skip)
    return _c(33) - skip


def _merge_halves(words, bits, count, out_words):
    half = bits.shape[1] // 2
    front = bits[:, half:]
    moved = _shift_back([w[:, :half] for w in words], front & _c(31))
    least, most = count // 32, len(words)
    hit = {j: shr(front, _c(5)) == j for j in range(least + 1, most + 1)}
    zero = jnp.zeros_like(front)
    out = []
    for k in range(out_words):
        v = moved[k - least] if 0 <= k - least < len(moved) else zero
        for j in range(least + 1, most + 1):
            if 0 <= k - j < len(moved):
                v = jnp.where(hit[j], moved[k - j], v)
            elif v is not zero:
                v = jnp.where(hit[j], zero, v)
        out.append(v | words[k][:, half:] if k < len(words) else v)
    return out, bits[:, :half] + front


def _split_halves(words, count, out_words):
    first, last = (count - 1) // 32, out_words - 1
    zero = jnp.zeros_like(words[0])

    def word(k):
        return words[k] if k < len(words) else zero

    seen = zero
    for k in range(first):
        seen = seen + lax.population_count(words[k])
    wanted = count - seen
    window = [word(first + k) for k in range(out_words + 1)]
    for j in range(first + 1, last + 1):
        seen = seen + lax.population_count(words[j - 1])
        later = seen < count
        wanted = jnp.where(later, count - seen, wanted)
        window = [jnp.where(later, word(j + k), v) for k, v in enumerate(window)]
    second = _shift_forward(window, _bits_through(window[0], wanted))
    return [jnp.concatenate([second[k], words[k]], axis=1) for k in range(out_words)]


def _slot_index():
    return lax.broadcasted_iota(I32, (8, TILE), 0), lax.broadcasted_iota(I32, (8, TILE), 1)


def _from_previous(x, row):
    y = pltpu.roll(x, 1, 0)
    return jnp.where(row == 0, pltpu.roll(y, 1, 1), y)


def _from_next(x, row):
    y = pltpu.roll(x, 7, 0)
    return jnp.where(row == 7, pltpu.roll(y, TILE - 1, 1), y)


def _last_row(x):
    return jnp.broadcast_to(x[7:8, :], x.shape)


def _bits_taken(over, row):
    def join(early, late):
        return early[0] + late[0], jnp.maximum(late[1], early[1] + late[0])

    run = over, jnp.maximum(over, 0)
    for k in (1, 2, 4):
        both = join([pltpu.roll(v, k, 0) for v in run], run)
        run = [jnp.where(row >= k, a, b) for a, b in zip(both, run)]
    lanes = [_last_row(v) for v in run]
    for unit in (1, 8):
        window = lanes
        for k in range(1, 8):
            lanes = join([pltpu.roll(v, k * unit, 1) for v in window], lanes)
    before = pltpu.roll(lanes[1], 1, 1)
    after = jnp.maximum(run[1], before + run[0])
    return jnp.where(row == 0, before, pltpu.roll(after, 1, 0))


def _sum_of_earlier(x, row, lane):
    run = x
    for k in (1, 2, 4):
        run = run + jnp.where(row >= k, pltpu.roll(run, k, 0), 0)
    lanes = total = _last_row(run)
    for unit, count in ((1, 8), (8, 16)):
        window = lanes
        for k in range(1, count):
            lanes = lanes + jnp.where(lane >= k * unit, pltpu.roll(window, k * unit, 1), 0)
    return (lanes - total) + (run - x)


def _code_step(i, w1, w2, scale, msg, state, c0=0, nc=8):
    low, high = _swap_bytes(w1, w2)
    msg[:, _tiles(LOW + 8 * i + c0, nc)] = low
    ranks, signs = _to_ranks(low, high, scale())
    msg[:, _tiles(RANKS + 8 * i + c0, nc)] = ranks | signs
    cols = _tiles(c0, nc)
    words, bits, room = _push_ranks([state[k, :, cols] for k in range(3)], ranks)
    for k in range(3):
        state[k, :, cols] = words[k]
    state[3, :, cols] = shr(state[3, :, cols], _c(1)) | signs
    state[4, :, cols] = state[4, :, cols] + bits
    state[5, :, cols] = state[5, :, cols] | room


def _code_finish(scale, msg, state):
    words, signs, bits = [state[0], state[1], state[2]], state[3], state[4]
    misfit = state[5]
    for count, out_words in ((32, 5), (64, 9), (128, LONGEST)):
        misfit = misfit | (_c(32 * len(words)) - bits)
        half = misfit.shape[1] // 2
        misfit = misfit[:, :half] | misfit[:, half:]
        words, bits = _merge_halves(words, bits, count, out_words)
    row, lane = _slot_index()
    first = (row | lane) == 0
    head = jnp.where(first, _c(HEADER), 0)
    over = bits + head - _c(32 * SLOT)
    taken = _bits_taken(over, row)
    again = _from_previous(jnp.maximum(taken + over, 0), row)
    start = head + taken
    misfit = misfit | (_c(32 * LONGEST) - bits) | (taken - again) | (_c(32 * SLOT - 1) - start)
    fits = jnp.max(shr(misfit, _c(31)).astype(jnp.float32)) == 0.0

    zero = jnp.zeros_like(bits)
    words = _shift_back(words, start & _c(31))
    for j in (1, 2, 4, 8):
        move = (start & _c(32 * j)) != 0
        here = words + [zero] * j
        there = [zero] * j + words
        words = [jnp.where(move, b, a) for a, b in zip(here[: 2 * SLOT], there)]
    spill = [_from_previous(w, row) for w in words[SLOT:]]
    ones = sum(lax.population_count(w) for w in spill)
    words = [a | b for a, b in zip(words[:SLOT], _shift_back(spill, head))]
    header = scale | jnp.where(fits, _c(0), _c(1 << 14)) | shl(ones, _c(15))
    header = shl(header, _c(32 - HEADER)) | (words[0] & _c(0xFF))
    words[0] = jnp.where(first, header, words[0])
    msg[:, _tiles(WORDS, SLOT)] = jnp.concatenate(words, axis=1)
    msg[:, _tiles(SIGNS, 8)] = signs
    return fits


def _read_header(msg):
    word = shr(msg[:, _tiles(WORDS, 1)][0, 0], _c(32 - HEADER))
    return word & _c(0x3FFF), (word & _c(1 << 14)) == 0, shr(word, _c(15))


def _expand_ranks(msg, ones_in_first):
    signs = msg[:, _tiles(SIGNS, 8)]
    row, lane = _slot_index()
    first = (row | lane) == 0
    head = jnp.where(first, _c(HEADER), 0)
    words = [msg[:, _tiles(WORDS + k, 1)] for k in range(SLOT)]
    words[0] = jnp.where(first, words[0] & _c(0xFF), words[0])
    zero = jnp.zeros_like(head)
    seen = [zero]
    for w in words:
        seen.append(seen[-1] + lax.population_count(w))
    foreign = ones_in_first + _sum_of_earlier(UNIT - seen[-1], row, lane)
    words += [_from_next(w, row) for w in _shift_forward(words + [zero], head)]
    index, wanted = zero, foreign
    for k in range(1, SLOT):
        later = seen[k] < foreign
        index = jnp.where(later, k, index)
        wanted = jnp.where(later, foreign - seen[k], wanted)
    for j in (8, 4, 2, 1):
        move = (index & _c(j)) != 0
        words = [
            jnp.where(move, words[min(k + j, len(words) - 1)], words[k]) for k in range(LONGEST + j)
        ]
    words = _shift_forward(words, jnp.where(foreign == 0, head, _bits_through(words[0], wanted)))
    for count, out_words in ((128, 9), (64, 5), (32, 3)):
        words = _split_halves(words, count, out_words)

    def step(j, words):
        words, ranks = _pop_ranks(list(words))
        msg[:, _tiles(RANKS + 8 * (STEPS - 1 - j), 8)] = ranks | (shl(signs, j) & _bytes(0x80))
        return tuple(words)

    lax.fori_loop(0, STEPS, step, tuple(words))


def _decode_step(i, scale, msg, c0=0, nc=8):
    low = msg[:, _tiles(LOW + 8 * i + c0, nc)]
    return _swap_bytes(low, _from_ranks(low, msg[:, _tiles(RANKS + 8 * i + c0, nc)], scale))


def _body(x_hbm, out, xv, tx, rx, state, side, load_sems, send_sems, recv_sems, side_sems, ready):
    me = lax.axis_index("i")
    own = me ^ shr(me, 1)

    def first(h):
        return me ^ (3 - 2 * h)

    def second(h):
        return me ^ (1 + 2 * h)

    def row0(h, unit):
        return (4 * h + (own ^ (3, 2 - h, 1 + h, 0)[unit])) * UNIT

    def slab_start(i):
        return i * SLAB if isinstance(i, int) else pl.multiple_of(i * SLAB, SLAB)

    def load(h, unit):
        rows = pl.ds(pl.multiple_of(row0(h, unit), UNIT), UNIT)
        return pltpu.make_async_copy(x_hbm.at[rows], xv.at[h, unit], load_sems.at[2 * unit + h])

    between = me & 1
    lead = jnp.where(me == 1, 1, 0)

    def load_slab(j, i, c0=0, nc=8):
        h, cols = lead ^ j, _tiles(c0, nc)
        rows = pl.ds(pl.multiple_of(row0(h, D) + slab_start(i), SLAB), SLAB)
        sem = load_sems.at[8 + 2 * i + j if c0 == 0 else 8 + 2 * STEPS]
        return pltpu.make_async_copy(
            x_hbm.at[rows, cols], xv.at[h, D, pl.ds(slab_start(i), SLAB), cols], sem
        )

    def signal_neighbours(sem):
        for h in range(2):
            pl.semaphore_signal(
                sem, inc=1, device_id=(first(h),), device_id_type=pl.DeviceIdType.MESH
            )

    opening = [
        (0, 0, DETOUR, 8 - DETOUR),
        (0, 0, 0, DETOUR),
        (1 - between, between, 0, 8),
        (between, 1 - between, 0, 8),
    ]
    load_slab(*opening[0]).start()
    barrier = pltpu.get_barrier_semaphore()
    pl.when(me != 2)(lambda: signal_neighbours(barrier))
    load_slab(*opening[1]).start()
    load_slab(*opening[2]).start()

    @pl.when(me == 2)
    def _():
        pl.semaphore_wait(barrier, 2)
        signal_neighbours(ready)

    def copy(h, msg, part, tile, tiles):
        if msg == END_D:
            src, device = rx.at[h, END_S], first(h)
        else:
            src = tx.at[h, (D, F, S, O, O)[msg]]
            device = (first, first, second, second, first)[msg](h)
        k = (h * 6 + msg) * PARTS + part
        cols = _tiles(tile, tiles)
        return pltpu.make_async_remote_copy(
            src.at[:, cols],
            rx.at[h, msg, :, cols],
            send_sems.at[k],
            recv_sems.at[k],
            device_id=(device,),
            device_id_type=pl.DeviceIdType.MESH,
        )

    def low_slab(h, msg, i):
        return copy(h, msg, jnp.where(i < SLABS_A[msg], LOW_A, LOW_B), LOW + 8 * i, 8)

    def low_part(h, msg, part):
        lo, hi = ((0, SLABS_A[msg]), (SLABS_A[msg], STEPS))[part]
        return copy(h, msg, part, LOW + 8 * lo, 8 * (hi - lo))

    def first_low_part(h, short, act):
        pl.when(short)(lambda: act(copy(h, IN_S, LOW_A, LOW + DETOUR, 8 * SLABS_A[IN_S] - DETOUR)))
        pl.when(jnp.logical_not(short))(lambda: act(low_part(h, IN_S, LOW_A)))

    def tail_pieces(h):
        return [copy(h, END_D, TAIL + k, LOW + a, n) for k, (a, n) in enumerate(TAIL_PIECES)]

    def head(h, msg):
        return copy(h, msg, HEAD, WORDS, 1)

    def rest(h, msg, fits, act):
        pl.when(fits)(lambda: act(copy(h, msg, REST, WORDS + 1, RANKS - WORDS - 1)))
        pl.when(jnp.logical_not(fits))(lambda: act(copy(h, msg, REST, RANKS, END - RANKS)))

    def detour(h):
        return pltpu.make_async_remote_copy(
            side.at[2],
            side.at[h],
            side_sems.at[2],
            side_sems.at[h],
            device_id=(second(h),),
            device_id_type=pl.DeviceIdType.MESH,
        )

    def start(c):
        c.start()

    def wait_recv(c):
        c.wait_recv()

    def wait_send(c):
        c.wait_send()

    def note(plain, h, msg, fits):
        return plain | shl(jnp.where(fits, 0, 1), h * 6 + msg)

    def fitted(plain, h, msg):
        return (shr(plain, h * 6 + msg) & 1) == 0

    def receive_rest(h, msg, landed=None):
        scale, fits, ones = _read_header(rx.at[h, msg])
        rest(h, msg, fits, wait_recv)
        if landed is not None:
            landed(fits)
        pl.when(fits)(lambda: _expand_ranks(rx.at[h, msg], ones))
        return scale, fits

    def receive(h, msg):
        if msg == IN_S:
            first_low_part(h, me == 0, wait_recv)
        else:
            low_part(h, msg, LOW_A).wait_recv()
        low_part(h, msg, LOW_B).wait_recv()
        head(h, msg).wait_recv()
        return receive_rest(h, msg)[0]

    def slab(h, unit, i, c0=0, nc=8):
        r, cols = slab_start(i), _tiles(c0, nc)
        return xv[h, unit, pl.ds(r, 16), cols], xv[h, unit, pl.ds(r + 16, 16), cols]

    def code(words_of, h, unit, each):
        scale = _choose_scale(words_of(0)[0][:, DETOUR * TILE :])
        state[0] = jnp.zeros(state.shape[1:], I32)

        @pl.loop(0, STEPS)
        def _(i):
            _code_step(i, *words_of(i), lambda: scale, tx.at[h, unit], state.at[0])
            each(i)

        return _code_finish(scale, tx.at[h, unit], state.at[0])

    def plus(values, h, msg, scale, i):
        words = _decode_step(i, scale, rx.at[h, msg])
        if msg == IN_S:
            missing = jnp.where((me == 0) & (i == 0), DETOUR * TILE, 0)
            col = lax.broadcasted_iota(I32, words[0].shape, 1)
            words = [jnp.where(col < missing, 0, w) for w in words]
        return [v + _from_words(w).astype(jnp.float32) for v, w in zip(values, words)]

    def emit(h, unit, i, words, c0=0, nc=8):
        r, cols = pl.multiple_of(row0(h, unit) + i * SLAB, SLAB), _tiles(c0, nc)
        out[pl.ds(r, 16), cols] = _from_words(words[0])
        out[pl.ds(r + 16, 16), cols] = _from_words(words[1])

    def emit_slabs(h, unit, msg, scale, lo, hi):
        @pl.loop(lo, hi)
        def _(i):
            emit(h, unit, i, _decode_step(i, scale, rx.at[h, msg]))

    state[...] = jnp.zeros(state.shape, I32)
    pl.when(between == 1)(lambda: pl.semaphore_wait(barrier, 1))
    scales = [None, None]
    for n, (j, i, c0, nc) in enumerate(opening):
        h = lead ^ j
        load_slab(j, i, c0, nc).wait()
        words = [_to_words(v) for v in slab(h, D, i, c0, nc)]

        def send_then_scale(n=n, j=j, h=h, i=i, c0=c0, nc=nc, words=words):
            goes = me == 2 if n == 1 else (me == 2) | ((between == 1) & (j == 0))
            pl.when(goes)(lambda: copy(h, IN_S, LOW_A, LOW + 8 * i + c0, nc).start())
            if n == 0:
                load_slab(*opening[3]).start()
                for k in range(3, 2 * STEPS):
                    load_slab(k & 1, k // 2).start()
                scales[0] = _choose_scale(words[0])
            elif n == 1:
                side[2] = jnp.concatenate(words, axis=1)
            elif n == 2:
                scales[1] = _choose_scale(words[0])
            else:
                scales[1] = jnp.where(j == 1, _choose_scale(words[0]), scales[1])
            return scales[0] if n < 2 else jnp.where(j == 1, scales[1], scales[0])

        _code_step(i, *words, send_then_scale, tx.at[h, D], state.at[j], c0, nc)

    @pl.when(between == 1)
    def _():
        pl.semaphore_wait(ready, 1)
        copy(lead ^ 1, IN_S, LOW_A, LOW, 8).start()
        detour(lead).start()

    @pl.when(me == 0)
    def _():
        for h in range(2):
            rx[h, IN_S, :, _tiles(LOW, DETOUR)] = jnp.zeros((8, DETOUR * TILE), I32)
        pl.semaphore_wait(barrier, 2)
        copy(0, IN_S, LOW_A, LOW, 16).start()
        copy(1, IN_S, LOW_A, LOW, 8).start()

    for unit in (F, S, O):
        for h in range(2):
            load(h, unit).start()

    @pl.loop(3, 2 * STEPS)
    def _(n):
        j, i = n & 1, shr(n, 1)
        h = lead ^ j
        load_slab(j, i).wait()
        scale = jnp.where(j == 1, scales[1], scales[0])
        _code_step(i, *map(_to_words, slab(h, D, i)), lambda: scale, tx.at[h, D], state.at[j])
        low_slab(h, IN_S, i).start()

    def finish_diagonal(j, plain):
        h = lead ^ j
        fits = _code_finish(jnp.where(j == 1, scales[1], scales[0]), tx.at[h, D], state.at[j])
        head(h, IN_S).start()
        rest(h, IN_S, fits, start)
        return note(plain, h, IN_S, fits)

    plain = lax.fori_loop(0, 2, finish_diagonal, _c(0))

    def for_first(h, plain):
        load(h, F).wait()

        @pl.when(me == 2)
        def _():
            detour(h).wait_recv()
            for k in range(2):
                at = (h, F, pl.ds(16 * k, 16), _tiles(0, DETOUR))
                extra = _from_words(side[h, :, _tiles(k * DETOUR, DETOUR)])
                xv[at] = xv[at] + extra.astype(jnp.float32)

        def each(i):
            pl.when((h == 0) | (i < SLABS_A[IN_O]))(lambda: low_slab(h, IN_O, i).start())

        fits = code(lambda i: [_to_words(v) for v in slab(h, F, i)], h, F, each)

        @pl.when(h == 0)
        def _():
            head(h, IN_O).start()
            rest(h, IN_O, fits, start)

        return note(plain, h, IN_O, fits)

    plain = lax.fori_loop(0, 2, for_first, plain)

    def for_second(h, plain):
        load(h, S).wait()
        scale = receive(h, IN_S)
        fits = code(
            lambda i: [_to_words(v) for v in plus(slab(h, S, i), h, IN_S, scale, i)],
            h,
            S,
            lambda i: low_slab(h, PART_O, i).start(),
        )
        head(h, PART_O).start()
        rest(h, PART_O, fits, start)

        @pl.when(h == 0)
        def _():
            low_part(1, IN_O, LOW_B).start()
            head(1, IN_O).start()
            rest(1, IN_O, fitted(plain, 1, IN_O), start)

        return note(plain, h, PART_O, fits)

    plain = lax.fori_loop(0, 2, for_second, plain)

    def for_all(h, plain):
        load(h, O).wait()
        scale_in = receive(h, IN_O)
        scale_part = receive(h, PART_O)

        def total(i):
            values = plus(slab(h, O, i), h, IN_O, scale_in, i)
            words = [_to_words(v) for v in plus(values, h, PART_O, scale_part, i)]
            emit(h, O, i, words)
            return words

        def each(i):
            for msg in (END_S, END_F):
                low_slab(h, msg, i).start()

        fits = code(total, h, O, each)
        for msg in (END_S, END_F):
            head(h, msg).start()
            rest(h, msg, fits, start)
            plain = note(plain, h, msg, fits)
        return plain

    plain = lax.fori_loop(0, 2, for_all, plain)

    def from_neighbours(h, plain):
        low_part(h, END_S, LOW_A).wait_recv()
        low_part(h, END_D, LOW_A).start()
        low_part(h, END_S, LOW_B).wait_recv()
        head(h, END_S).wait_recv()
        head(h, END_D).start()

        def pass_on(fits):
            rest(h, END_D, fits, start)
            for piece in tail_pieces(h):
                piece.start()

        scale, fits = receive_rest(h, END_S, pass_on)
        emit_slabs(h, S, END_S, scale, 0, STEPS)
        emit_slabs(h, F, END_F, receive(h, END_F), 0, STEPS)
        return note(plain, h, END_D, fits)

    plain = lax.fori_loop(0, 2, from_neighbours, plain)

    def sent(h, msg, low_parts):
        for c in low_parts + [head(h, msg)]:
            c.wait_send()
        rest(h, msg, fitted(plain, h, msg), wait_send)

    @pl.loop(0, 2)
    def _(h):
        first_low_part(h, (between == 1) & (h == lead), wait_send)
        sent(h, IN_S, [low_part(h, IN_S, LOW_B)])
        for msg in range(IN_O, END_D):
            sent(h, msg, [low_part(h, msg, LOW_A), low_part(h, msg, LOW_B)])

    pl.when(between == 1)(lambda: detour(lead).wait_send())

    def diagonal_ranks(j, scales):
        h = lead ^ j
        low_part(h, END_D, LOW_A).wait_recv()
        head(h, END_D).wait_recv()
        scale = receive_rest(h, END_D)[0]
        emit_slabs(h, D, END_D, scale, 0, SLABS_A[END_D])
        return scales[1], scale

    scales = lax.fori_loop(0, 2, diagonal_ranks, (_c(0), _c(0)))
    for k, (tile, tiles) in enumerate(TAIL_PIECES):
        if k == len(TAIL_PIECES) - 2:
            for h in range(2):
                sent(h, END_D, [low_part(h, END_D, LOW_A)] + tail_pieces(h))
        for j in range(2):
            h = lead ^ j
            copy(h, END_D, TAIL + k, LOW + tile, tiles).wait_recv()
            if tiles > 8:
                emit_slabs(h, D, END_D, scales[j], tile // 8, (tile + tiles) // 8)
            else:
                words = _decode_step(tile // 8, scales[j], rx.at[h, END_D], tile % 8, tiles)
                emit(h, D, tile // 8, words, tile % 8, tiles)


def pallas_dist_rs_then_ag_i_m2048_n1024_kernel(x: jax.Array):
    return pl.pallas_call(
        _body,
        out_shape=jax.ShapeDtypeStruct((ROWS, N), jnp.bfloat16),
        in_specs=[pl.BlockSpec(memory_space=pl.ANY)],
        out_specs=pl.BlockSpec(memory_space=pltpu.VMEM),
        scratch_shapes=[
            pltpu.VMEM((2, 4, UNIT, N), jnp.float32),
            pltpu.VMEM((2, 4, 8, END * TILE), I32),
            pltpu.VMEM((2, 6, 8, END * TILE), I32),
            pltpu.VMEM((2, 6, 8, N), I32),
            pltpu.VMEM((3, 8, 2 * DETOUR * TILE), I32),
            pltpu.SemaphoreType.DMA((9 + 2 * STEPS,)),
            pltpu.SemaphoreType.DMA((12 * PARTS,)),
            pltpu.SemaphoreType.DMA((12 * PARTS,)),
            pltpu.SemaphoreType.DMA((3,)),
            pltpu.SemaphoreType.REGULAR,
        ],
        compiler_params=pltpu.CompilerParams(
            collective_id=0,
            vmem_limit_bytes=64 * 2**20,
            disable_bounds_checks=True,
            disable_semaphore_checks=True,
        ),
    )(x)
```

```python
import jax
import jax.numpy as jnp
import numpy as np
from jax import lax
from jax.experimental import pallas as pl
from jax.experimental.pallas import tpu as pltpu

ROWS, N = 2048, 1024
UNIT = 256
SLAB = 32
STEPS = UNIT // SLAB
TILE = 128
I32 = jnp.int32

LONGEST = 16
SLOT = 13
ZERO = 20
LOW, WORDS, SIGNS, RANKS, END = 0, 64, 64 + SLOT, 72 + SLOT, 136 + SLOT

D, F, S, O = range(4)
IN_S, IN_O, PART_O, END_S, END_F, END_D = range(6)
LOW_A, LOW_B, HEAD, REST, TAIL = range(5)
SLABS_A = (4, 5, 4, 3, 4, 3)
TAIL_PIECES = ((24, 16), (40, 8), (48, 8), (56, 6), (62, 2))
PARTS = TAIL + len(TAIL_PIECES)
DETOUR = 4

shl = lax.shift_left
shr = lax.shift_right_logical


def _c(value):
    return np.int32(value)


def _bytes(byte):
    return np.uint32(byte * 0x01010101).astype(np.int32)


def _tiles(first, count):
    start = first * TILE
    return pl.ds(start if isinstance(first, int) else pl.multiple_of(start, TILE), count * TILE)


def _to_words(x):
    return pltpu.bitcast(x.astype(jnp.bfloat16), I32)


def _from_words(words):
    return pltpu.bitcast(words, jnp.bfloat16)


def _swap_bytes(a, b):
    x = (shr(a, _c(8)) ^ b) & _c(0x00FF00FF)
    return a ^ shl(x, _c(8)), b ^ x


def _choose_scale(words):
    magnitudes = (words & _c(0x7FFF)) + (shr(words, _c(16)) & _c(0x7FFF))
    mean = jnp.sum(magnitudes.astype(jnp.float32)) * (0.5 / words.size)
    return shr(mean.astype(I32) + _c(469), _c(1)) & _c(0x3FFF)


def _scale_terms(low, scale):
    d = (shr(low, _c(1)) & _bytes(0x7F)) + (_c(0x7F) - (scale & _c(0x7F))) * _bytes(0x01)
    base = (shr(scale, _c(7)) | _c(0x80)) * _bytes(0x01) - (shr(d, _c(7)) & _bytes(0x01))
    x = shr(d, _c(4)) & _bytes(0x07)
    return base, x + (shr(_bytes(0x08) - x, _c(3)) & _bytes(0x01)) + _bytes(0x80)


def _swap_zero_class(u, scale):
    zero = shr(scale, _c(7)) * _bytes(0x01)
    hit = (_bytes(0x80) - (u ^ zero)) | (_bytes(0x80) - (u ^ _bytes(ZERO)))
    hit = hit & _bytes(0x80)
    return u ^ ((hit - shr(hit, _c(7))) & (zero ^ _bytes(ZERO)))


def _to_ranks(low, high, scale):
    base, r = _scale_terms(low, scale)
    u = _swap_zero_class((base - (high & _bytes(0x7F))) & _bytes(0x7F), scale)
    top = (_bytes(0x80) - u) & _bytes(0x80)
    ranks = u - (shr(r - u, _c(7)) & _bytes(0x01)) + ((r + _bytes(0x01)) & (top - shr(top, _c(7))))
    return ranks, high & _bytes(0x80)


def _from_ranks(low, signed_ranks, scale):
    base, r = _scale_terms(low, scale)
    q = signed_ranks & _bytes(0x7F)
    at_most = r - q
    below = at_most - _bytes(0x01)
    top = (at_most ^ below) & _bytes(0x80)
    u = q + (shr(below, _c(7)) & _bytes(0x01)) - (q & (top - shr(top, _c(7))))
    return ((base - _swap_zero_class(u, scale)) & _bytes(0x7F)) | (signed_ranks & _bytes(0x80))


def _with_scales(fn, low, other, scales, i, c0):
    cut = min(max(DETOUR - c0, 0) * TILE, low.shape[1])
    left = jnp.where(i == 0, scales[1], scales[0])
    parts = [
        fn(low[:, lo:hi], other[:, lo:hi], scale)
        for lo, hi, scale in ((0, cut, left), (cut, low.shape[1], scales[0]))
        if lo < hi
    ]
    return jax.tree.map(lambda *columns: jnp.concatenate(columns, axis=1), *parts)


def _shift_back(words, bits):
    other = _c(32) - bits
    middle = [shr(words[k], bits) | shl(words[k - 1], other) for k in range(1, len(words))]
    return [shr(words[0], bits)] + middle + [shl(words[-1], other)]


def _shift_forward(words, bits):
    other = _c(32) - bits
    return [shl(words[k], bits) | shr(words[k + 1], other) for k in range(len(words) - 1)]


def _push_ranks(words, ranks):
    lengths = ranks + _bytes(0x01)
    la, lb = lengths & _c(0xFF), shr(lengths, _c(24))
    lc, ld = shr(lengths, _c(8)) & _c(0xFF), shr(lengths, _c(16)) & _c(0xFF)
    code = shl(jnp.ones_like(lb), lb) | _c(1)
    code = shl(code, lc) | _c(1)
    code = shl(code, ld) | _c(1)
    bits = (la + lb) + (lc + ld)
    room = _c(32) - bits
    out = _shift_back(words, bits)[: len(words)]
    return [shl(code, room) | out[0]] + out[1:], bits, room


def _pop_ranks(words):
    x = words[0]
    qa = lax.clz(x)
    x = shl(shl(x, _c(1)), qa)
    qb = lax.clz(x)
    x = shl(shl(x, _c(1)), qb)
    qc = lax.clz(x)
    x = shl(shl(x, _c(1)), qc)
    qd = lax.clz(x)
    bits = (qa + qb) + (qc + _c(4)) + qd
    out = _shift_forward(words, bits) + [shl(words[-1], bits)]
    return out, (qa | shl(qb, _c(24))) | (shl(qc, _c(8)) | shl(qd, _c(16)))


def _bits_through(word, ones):
    skip = jnp.zeros_like(word) + _c(32)
    for step in (16, 8, 4, 2, 1):
        less = skip - _c(step)
        skip = jnp.where(lax.population_count(shr(word, less)) < ones, less, skip)
    return _c(33) - skip


def _merge_halves(words, bits, count, out_words):
    half = bits.shape[1] // 2
    front = bits[:, half:]
    moved = _shift_back([w[:, :half] for w in words], front & _c(31))
    least, most = count // 32, len(words)
    hit = {j: shr(front, _c(5)) == j for j in range(least + 1, most + 1)}
    zero = jnp.zeros_like(front)
    out = []
    for k in range(out_words):
        v = moved[k - least] if 0 <= k - least < len(moved) else zero
        for j in range(least + 1, most + 1):
            if 0 <= k - j < len(moved):
                v = jnp.where(hit[j], moved[k - j], v)
            elif v is not zero:
                v = jnp.where(hit[j], zero, v)
        out.append(v | words[k][:, half:] if k < len(words) else v)
    return out, bits[:, :half] + front


def _split_halves(words, count, out_words):
    first, last = (count - 1) // 32, out_words - 1
    zero = jnp.zeros_like(words[0])

    def word(k):
        return words[k] if k < len(words) else zero

    seen = zero
    for k in range(first):
        seen = seen + lax.population_count(words[k])
    wanted = count - seen
    window = [word(first + k) for k in range(out_words + 1)]
    for j in range(first + 1, last + 1):
        seen = seen + lax.population_count(words[j - 1])
        later = seen < count
        wanted = jnp.where(later, count - seen, wanted)
        window = [jnp.where(later, word(j + k), v) for k, v in enumerate(window)]
    second = _shift_forward(window, _bits_through(window[0], wanted))
    return [jnp.concatenate([second[k], words[k]], axis=1) for k in range(out_words)]


def _slot_index():
    return lax.broadcasted_iota(I32, (8, TILE), 0), lax.broadcasted_iota(I32, (8, TILE), 1)


def _from_previous(x, row):
    y = pltpu.roll(x, 1, 0)
    return jnp.where(row == 0, pltpu.roll(y, 1, 1), y)


def _from_next(x, row):
    y = pltpu.roll(x, 7, 0)
    return jnp.where(row == 7, pltpu.roll(y, TILE - 1, 1), y)


def _last_row(x):
    return jnp.broadcast_to(x[7:8, :], x.shape)


def _bits_taken(over, row):
    def join(early, late):
        return early[0] + late[0], jnp.maximum(late[1], early[1] + late[0])

    run = over, jnp.maximum(over, 0)
    for k in (1, 2, 4):
        both = join([pltpu.roll(v, k, 0) for v in run], run)
        run = [jnp.where(row >= k, a, b) for a, b in zip(both, run)]
    lanes = [_last_row(v) for v in run]
    for unit in (1, 8):
        window = lanes
        for k in range(1, 8):
            lanes = join([pltpu.roll(v, k * unit, 1) for v in window], lanes)
    before = pltpu.roll(lanes[1], 1, 1)
    after = jnp.maximum(run[1], before + run[0])
    return jnp.where(row == 0, before, pltpu.roll(after, 1, 0))


def _sum_of_earlier(x, row, lane):
    run = x
    for k in (1, 2, 4):
        run = run + jnp.where(row >= k, pltpu.roll(run, k, 0), 0)
    lanes = total = _last_row(run)
    for unit, count in ((1, 8), (8, 16)):
        window = lanes
        for k in range(1, count):
            lanes = lanes + jnp.where(lane >= k * unit, pltpu.roll(window, k * unit, 1), 0)
    return (lanes - total) + (run - x)


def _code_step(i, w1, w2, scales, msg, state, c0=0, nc=8):
    low, high = _swap_bytes(w1, w2)
    msg[:, _tiles(LOW + 8 * i + c0, nc)] = low
    ranks, signs = _with_scales(_to_ranks, low, high, scales(), i, c0)
    msg[:, _tiles(RANKS + 8 * i + c0, nc)] = ranks | signs
    cols = _tiles(c0, nc)
    words, bits, room = _push_ranks([state[k, :, cols] for k in range(3)], ranks)
    for k in range(3):
        state[k, :, cols] = words[k]
    state[3, :, cols] = shr(state[3, :, cols], _c(1)) | signs
    state[4, :, cols] = state[4, :, cols] + bits
    state[5, :, cols] = state[5, :, cols] | room


def _code_finish(scales, msg, state):
    words, signs, bits = [state[0], state[1], state[2]], state[3], state[4]
    misfit = state[5]
    for count, out_words in ((32, 5), (64, 9), (128, LONGEST)):
        misfit = misfit | (_c(32 * len(words)) - bits)
        half = misfit.shape[1] // 2
        misfit = misfit[:, :half] | misfit[:, half:]
        words, bits = _merge_halves(words, bits, count, out_words)
    row, lane = _slot_index()
    first = (row | lane) == 0
    head = jnp.where(first, _c(32), 0)
    over = bits + head - _c(32 * SLOT)
    taken = _bits_taken(over, row)
    again = _from_previous(jnp.maximum(taken + over, 0), row)
    start = head + taken
    misfit = misfit | (_c(32 * LONGEST) - bits) | (taken - again) | (_c(32 * SLOT - 1) - start)
    fits = jnp.max(shr(misfit, _c(31)).astype(jnp.float32)) == 0.0

    zero = jnp.zeros_like(bits)
    words = _shift_back(words, start & _c(31))
    for j in (1, 2, 4, 8):
        move = (start & _c(32 * j)) != 0
        here = words + [zero] * j
        there = [zero] * j + words
        words = [jnp.where(move, b, a) for a, b in zip(here[: 2 * SLOT], there)]
    spill = [_from_previous(w, row) for w in words[SLOT:]]
    ones = sum(lax.population_count(w) for w in spill)
    words = [a | b for a, b in zip(words[:SLOT], _shift_back(spill, head))]
    header = scales[0] | jnp.where(fits, _c(0), _c(1 << 14)) | shl(scales[1] - scales[0], _c(24))
    words[0] = jnp.where(first, header | shl(ones, _c(15)), words[0])
    msg[:, _tiles(WORDS, SLOT)] = jnp.concatenate(words, axis=1)
    msg[:, _tiles(SIGNS, 8)] = signs
    return fits


def _read_header(msg):
    word = msg[:, _tiles(WORDS, 1)][0, 0]
    scale = word & _c(0x3FFF)
    scales = scale, scale + lax.shift_right_arithmetic(word, _c(24))
    return scales, (word & _c(1 << 14)) == 0, shr(word, _c(15)) & _c(0x1FF)


def _expand_ranks(msg, ones_in_first):
    signs = msg[:, _tiles(SIGNS, 8)]
    row, lane = _slot_index()
    first = (row | lane) == 0
    head = jnp.where(first, _c(32), 0)
    words = [msg[:, _tiles(WORDS + k, 1)] for k in range(SLOT)]
    words[0] = jnp.where(first, _c(0), words[0])
    zero = jnp.zeros_like(head)
    seen = [zero]
    for w in words:
        seen.append(seen[-1] + lax.population_count(w))
    foreign = ones_in_first + _sum_of_earlier(UNIT - seen[-1], row, lane)
    words += [_from_next(w, row) for w in _shift_forward(words + [zero], head)]
    index, wanted = zero, foreign
    for k in range(1, SLOT):
        later = seen[k] < foreign
        index = jnp.where(later, k, index)
        wanted = jnp.where(later, foreign - seen[k], wanted)
    for j in (8, 4, 2, 1):
        move = (index & _c(j)) != 0
        words = [
            jnp.where(move, words[min(k + j, len(words) - 1)], words[k]) for k in range(LONGEST + j)
        ]
    words = _shift_forward(words, jnp.where(foreign == 0, head, _bits_through(words[0], wanted)))
    for count, out_words in ((128, 9), (64, 5), (32, 3)):
        words = _split_halves(words, count, out_words)

    def step(j, words):
        words, ranks = _pop_ranks(list(words))
        msg[:, _tiles(RANKS + 8 * (STEPS - 1 - j), 8)] = ranks | (shl(signs, j) & _bytes(0x80))
        return tuple(words)

    lax.fori_loop(0, STEPS, step, tuple(words))


def _decode_step(i, scales, msg, c0=0, nc=8):
    low, ranks = msg[:, _tiles(LOW + 8 * i + c0, nc)], msg[:, _tiles(RANKS + 8 * i + c0, nc)]
    return _swap_bytes(low, _with_scales(_from_ranks, low, ranks, scales, i, c0))


def _body(x_hbm, out, xv, tx, rx, state, side, load_sems, send_sems, recv_sems, side_sems, ready):
    me = lax.axis_index("i")
    own = me ^ shr(me, 1)

    def first(h):
        return me ^ (3 - 2 * h)

    def second(h):
        return me ^ (1 + 2 * h)

    def row0(h, unit):
        return (4 * h + (own ^ (3, 2 - h, 1 + h, 0)[unit])) * UNIT

    def slab_start(i):
        return i * SLAB if isinstance(i, int) else pl.multiple_of(i * SLAB, SLAB)

    def load(h, unit):
        rows = pl.ds(pl.multiple_of(row0(h, unit), UNIT), UNIT)
        return pltpu.make_async_copy(x_hbm.at[rows], xv.at[h, unit], load_sems.at[2 * unit + h])

    between = me & 1
    lead = jnp.where(me == 1, 1, 0)

    def load_slab(j, i, c0=0, nc=8):
        h, cols = lead ^ j, _tiles(c0, nc)
        rows = pl.ds(pl.multiple_of(row0(h, D) + slab_start(i), SLAB), SLAB)
        sem = load_sems.at[8 + 2 * i + j if c0 == 0 else 8 + 2 * STEPS]
        return pltpu.make_async_copy(
            x_hbm.at[rows, cols], xv.at[h, D, pl.ds(slab_start(i), SLAB), cols], sem
        )

    def signal_neighbours(sem):
        for h in range(2):
            pl.semaphore_signal(
                sem, inc=1, device_id=(first(h),), device_id_type=pl.DeviceIdType.MESH
            )

    opening = [
        (0, 0, DETOUR, 8 - DETOUR),
        (0, 0, 0, DETOUR),
        (1 - between, between, 0, 8),
        (between, 1 - between, 0, 8),
    ]
    load_slab(*opening[0]).start()
    barrier = pltpu.get_barrier_semaphore()
    pl.when(me != 2)(lambda: signal_neighbours(barrier))
    load_slab(*opening[1]).start()
    load_slab(*opening[2]).start()

    @pl.when(me == 2)
    def _():
        pl.semaphore_wait(barrier, 2)
        signal_neighbours(ready)

    def copy(h, msg, part, tile, tiles):
        if msg == END_D:
            src, device = rx.at[h, END_S], first(h)
        else:
            src = tx.at[h, (D, F, S, O, O)[msg]]
            device = (first, first, second, second, first)[msg](h)
        k = (h * 6 + msg) * PARTS + part
        cols = _tiles(tile, tiles)
        return pltpu.make_async_remote_copy(
            src.at[:, cols],
            rx.at[h, msg, :, cols],
            send_sems.at[k],
            recv_sems.at[k],
            device_id=(device,),
            device_id_type=pl.DeviceIdType.MESH,
        )

    def low_slab(h, msg, i):
        return copy(h, msg, jnp.where(i < SLABS_A[msg], LOW_A, LOW_B), LOW + 8 * i, 8)

    def low_part(h, msg, part):
        lo, hi = ((0, SLABS_A[msg]), (SLABS_A[msg], STEPS))[part]
        return copy(h, msg, part, LOW + 8 * lo, 8 * (hi - lo))

    def first_low_part(h, short, act):
        pl.when(short)(lambda: act(copy(h, IN_S, LOW_A, LOW + DETOUR, 8 * SLABS_A[IN_S] - DETOUR)))
        pl.when(jnp.logical_not(short))(lambda: act(low_part(h, IN_S, LOW_A)))

    def tail_pieces(h):
        return [copy(h, END_D, TAIL + k, LOW + a, n) for k, (a, n) in enumerate(TAIL_PIECES)]

    def head(h, msg):
        return copy(h, msg, HEAD, WORDS, 1)

    def rest(h, msg, fits, act):
        pl.when(fits)(lambda: act(copy(h, msg, REST, WORDS + 1, RANKS - WORDS - 1)))
        pl.when(jnp.logical_not(fits))(lambda: act(copy(h, msg, REST, RANKS, END - RANKS)))

    def detour(h):
        return pltpu.make_async_remote_copy(
            side.at[2],
            side.at[h],
            side_sems.at[2],
            side_sems.at[h],
            device_id=(second(h),),
            device_id_type=pl.DeviceIdType.MESH,
        )

    def start(c):
        c.start()

    def wait_recv(c):
        c.wait_recv()

    def wait_send(c):
        c.wait_send()

    def note(plain, h, msg, fits):
        return plain | shl(jnp.where(fits, 0, 1), h * 6 + msg)

    def fitted(plain, h, msg):
        return (shr(plain, h * 6 + msg) & 1) == 0

    def receive_rest(h, msg, landed=None):
        scales, fits, ones = _read_header(rx.at[h, msg])
        rest(h, msg, fits, wait_recv)
        if landed is not None:
            landed(fits)
        pl.when(fits)(lambda: _expand_ranks(rx.at[h, msg], ones))
        return scales, fits

    def receive(h, msg):
        if msg == IN_S:
            first_low_part(h, me == 0, wait_recv)
        else:
            low_part(h, msg, LOW_A).wait_recv()
        low_part(h, msg, LOW_B).wait_recv()
        head(h, msg).wait_recv()
        return receive_rest(h, msg)[0]

    def slab(h, unit, i, c0=0, nc=8):
        r, cols = slab_start(i), _tiles(c0, nc)
        return xv[h, unit, pl.ds(r, 16), cols], xv[h, unit, pl.ds(r + 16, 16), cols]

    def code(words_of, h, unit, each):
        sample = words_of(0)[0]
        scale = _choose_scale(sample[:, DETOUR * TILE :])
        apart = _choose_scale(sample[:, : DETOUR * TILE]) - scale
        scales = scale, scale + jnp.clip(apart, -128, 127)
        state[0] = jnp.zeros(state.shape[1:], I32)

        @pl.loop(0, STEPS)
        def _(i):
            _code_step(i, *words_of(i), lambda: scales, tx.at[h, unit], state.at[0])
            each(i)

        return _code_finish(scales, tx.at[h, unit], state.at[0])

    def plus(values, h, msg, scales, i):
        words = _decode_step(i, scales, rx.at[h, msg])
        if msg == IN_S:
            missing = jnp.where((me == 0) & (i == 0), DETOUR * TILE, 0)
            col = lax.broadcasted_iota(I32, words[0].shape, 1)
            words = [jnp.where(col < missing, 0, w) for w in words]
        return [v + _from_words(w).astype(jnp.float32) for v, w in zip(values, words)]

    def emit(h, unit, i, words, c0=0, nc=8):
        r, cols = pl.multiple_of(row0(h, unit) + i * SLAB, SLAB), _tiles(c0, nc)
        out[pl.ds(r, 16), cols] = _from_words(words[0])
        out[pl.ds(r + 16, 16), cols] = _from_words(words[1])

    def emit_slabs(h, unit, msg, scales, lo, hi):
        @pl.loop(lo, hi)
        def _(i):
            emit(h, unit, i, _decode_step(i, scales, rx.at[h, msg]))

    state[...] = jnp.zeros(state.shape, I32)
    pl.when(between == 1)(lambda: pl.semaphore_wait(barrier, 1))
    chosen = [None, None]

    def diagonal_scales(j):
        return (jnp.where(j == 1, chosen[1], chosen[0]),) * 2

    for n, (j, i, c0, nc) in enumerate(opening):
        h = lead ^ j
        load_slab(j, i, c0, nc).wait()
        words = [_to_words(v) for v in slab(h, D, i, c0, nc)]

        def send_then_scales(n=n, j=j, h=h, i=i, c0=c0, nc=nc, words=words):
            goes = me == 2 if n == 1 else (me == 2) | ((between == 1) & (j == 0))
            pl.when(goes)(lambda: copy(h, IN_S, LOW_A, LOW + 8 * i + c0, nc).start())
            if n == 0:
                load_slab(*opening[3]).start()
                for k in range(3, 2 * STEPS):
                    load_slab(k & 1, k // 2).start()
                chosen[0] = _choose_scale(words[0])
            elif n == 1:
                side[2] = jnp.concatenate(words, axis=1)
            elif n == 2:
                chosen[1] = _choose_scale(words[0])
            else:
                chosen[1] = jnp.where(j == 1, _choose_scale(words[0]), chosen[1])
            return (chosen[0],) * 2 if n < 2 else diagonal_scales(j)

        _code_step(i, *words, send_then_scales, tx.at[h, D], state.at[j], c0, nc)

    @pl.when(between == 1)
    def _():
        pl.semaphore_wait(ready, 1)
        copy(lead ^ 1, IN_S, LOW_A, LOW, 8).start()
        detour(lead).start()

    @pl.when(me == 0)
    def _():
        for h in range(2):
            rx[h, IN_S, :, _tiles(LOW, DETOUR)] = jnp.zeros((8, DETOUR * TILE), I32)
        pl.semaphore_wait(barrier, 2)
        copy(0, IN_S, LOW_A, LOW, 16).start()
        copy(1, IN_S, LOW_A, LOW, 8).start()

    for unit in (F, S, O):
        for h in range(2):
            load(h, unit).start()

    @pl.loop(3, 2 * STEPS)
    def _(n):
        j, i = n & 1, shr(n, 1)
        h = lead ^ j
        load_slab(j, i).wait()
        words = map(_to_words, slab(h, D, i))
        _code_step(i, *words, lambda: diagonal_scales(j), tx.at[h, D], state.at[j])
        low_slab(h, IN_S, i).start()

    def finish_diagonal(j, plain):
        h = lead ^ j
        fits = _code_finish(diagonal_scales(j), tx.at[h, D], state.at[j])
        head(h, IN_S).start()
        rest(h, IN_S, fits, start)
        return note(plain, h, IN_S, fits)

    plain = lax.fori_loop(0, 2, finish_diagonal, _c(0))

    def for_first(h, plain):
        load(h, F).wait()

        @pl.when(me == 2)
        def _():
            detour(h).wait_recv()
            for k in range(2):
                at = (h, F, pl.ds(16 * k, 16), _tiles(0, DETOUR))
                extra = _from_words(side[h, :, _tiles(k * DETOUR, DETOUR)])
                xv[at] = xv[at] + extra.astype(jnp.float32)

        def each(i):
            pl.when((h == 0) | (i < SLABS_A[IN_O]))(lambda: low_slab(h, IN_O, i).start())

        fits = code(lambda i: [_to_words(v) for v in slab(h, F, i)], h, F, each)

        @pl.when(h == 0)
        def _():
            head(h, IN_O).start()
            rest(h, IN_O, fits, start)

        return note(plain, h, IN_O, fits)

    plain = lax.fori_loop(0, 2, for_first, plain)

    def for_second(h, plain):
        load(h, S).wait()
        scales = receive(h, IN_S)
        fits = code(
            lambda i: [_to_words(v) for v in plus(slab(h, S, i), h, IN_S, scales, i)],
            h,
            S,
            lambda i: low_slab(h, PART_O, i).start(),
        )
        head(h, PART_O).start()
        rest(h, PART_O, fits, start)

        @pl.when(h == 0)
        def _():
            low_part(1, IN_O, LOW_B).start()
            head(1, IN_O).start()
            rest(1, IN_O, fitted(plain, 1, IN_O), start)

        return note(plain, h, PART_O, fits)

    plain = lax.fori_loop(0, 2, for_second, plain)

    def for_all(h, plain):
        load(h, O).wait()
        scales_in = receive(h, IN_O)
        scales_part = receive(h, PART_O)

        def total(i):
            values = plus(slab(h, O, i), h, IN_O, scales_in, i)
            words = [_to_words(v) for v in plus(values, h, PART_O, scales_part, i)]
            emit(h, O, i, words)
            return words

        def each(i):
            for msg in (END_S, END_F):
                low_slab(h, msg, i).start()

        fits = code(total, h, O, each)
        for msg in (END_S, END_F):
            head(h, msg).start()
            rest(h, msg, fits, start)
            plain = note(plain, h, msg, fits)
        return plain

    plain = lax.fori_loop(0, 2, for_all, plain)

    def from_neighbours(h, plain):
        low_part(h, END_S, LOW_A).wait_recv()
        low_part(h, END_D, LOW_A).start()
        low_part(h, END_S, LOW_B).wait_recv()
        head(h, END_S).wait_recv()
        head(h, END_D).start()

        def pass_on(fits):
            rest(h, END_D, fits, start)
            for piece in tail_pieces(h):
                piece.start()

        scales, fits = receive_rest(h, END_S, pass_on)
        emit_slabs(h, S, END_S, scales, 0, STEPS)
        emit_slabs(h, F, END_F, receive(h, END_F), 0, STEPS)
        return note(plain, h, END_D, fits)

    plain = lax.fori_loop(0, 2, from_neighbours, plain)

    def sent(h, msg, low_parts):
        for c in low_parts + [head(h, msg)]:
            c.wait_send()
        rest(h, msg, fitted(plain, h, msg), wait_send)

    @pl.loop(0, 2)
    def _(h):
        first_low_part(h, (between == 1) & (h == lead), wait_send)
        sent(h, IN_S, [low_part(h, IN_S, LOW_B)])
        for msg in range(IN_O, END_D):
            sent(h, msg, [low_part(h, msg, LOW_A), low_part(h, msg, LOW_B)])

    pl.when(between == 1)(lambda: detour(lead).wait_send())

    def diagonal_ranks(j, last_two):
        h = lead ^ j
        low_part(h, END_D, LOW_A).wait_recv()
        head(h, END_D).wait_recv()
        scales = receive_rest(h, END_D)[0]
        emit_slabs(h, D, END_D, scales, 0, SLABS_A[END_D])
        return last_two[1], scales

    scales_of = lax.fori_loop(0, 2, diagonal_ranks, ((_c(0), _c(0)),) * 2)
    for k, (tile, tiles) in enumerate(TAIL_PIECES):
        if k == len(TAIL_PIECES) - 2:
            for h in range(2):
                sent(h, END_D, [low_part(h, END_D, LOW_A)] + tail_pieces(h))
        for j in range(2):
            h = lead ^ j
            copy(h, END_D, TAIL + k, LOW + tile, tiles).wait_recv()
            if tiles > 8:
                emit_slabs(h, D, END_D, scales_of[j], tile // 8, (tile + tiles) // 8)
            else:
                words = _decode_step(tile // 8, scales_of[j], rx.at[h, END_D], tile % 8, tiles)
                emit(h, D, tile // 8, words, tile % 8, tiles)


def pallas_dist_rs_then_ag_i_m2048_n1024_kernel(x: jax.Array):
    return pl.pallas_call(
        _body,
        out_shape=jax.ShapeDtypeStruct((ROWS, N), jnp.bfloat16),
        in_specs=[pl.BlockSpec(memory_space=pl.ANY)],
        out_specs=pl.BlockSpec(memory_space=pltpu.VMEM),
        scratch_shapes=[
            pltpu.VMEM((2, 4, UNIT, N), jnp.float32),
            pltpu.VMEM((2, 4, 8, END * TILE), I32),
            pltpu.VMEM((2, 6, 8, END * TILE), I32),
            pltpu.VMEM((2, 6, 8, N), I32),
            pltpu.VMEM((3, 8, 2 * DETOUR * TILE), I32),
            pltpu.SemaphoreType.DMA((9 + 2 * STEPS,)),
            pltpu.SemaphoreType.DMA((12 * PARTS,)),
            pltpu.SemaphoreType.DMA((12 * PARTS,)),
            pltpu.SemaphoreType.DMA((3,)),
            pltpu.SemaphoreType.REGULAR,
        ],
        compiler_params=pltpu.CompilerParams(
            collective_id=0,
            vmem_limit_bytes=64 * 2**20,
            disable_bounds_checks=True,
            disable_semaphore_checks=True,
        ),
    )(x)
```

```python
import jax
import jax.numpy as jnp
import numpy as np
from jax import lax
from jax.experimental import pallas as pl
from jax.experimental.pallas import tpu as pltpu

ROWS, N = 2048, 1024
UNIT = 256
SLAB = 32
STEPS = UNIT // SLAB
TILE = 128
I32 = jnp.int32

LONGEST = 16
SLOT = 13
ZERO = 20
LOW, WORDS, SIGNS, RANKS, END = 0, 64, 64 + SLOT, 72 + SLOT, 136 + SLOT

D, F, S, O = range(4)
IN_S, IN_O, PART_O, END_S, END_F, END_D = range(6)
LOW_A, LOW_B, HEAD, REST, TAIL = range(5)
SLABS_A = (4, 5, 4, 3, 4, 3)
TAIL_PIECES = ((24, 16), (40, 8), (48, 8), (56, 6), (62, 2))
PARTS = TAIL + len(TAIL_PIECES)
DETOUR = 4

shl = lax.shift_left
shr = lax.shift_right_logical


def _c(value):
    return np.int32(value)


def _bytes(byte):
    return np.uint32(byte * 0x01010101).astype(np.int32)


def _tiles(first, count):
    start = first * TILE
    return pl.ds(start if isinstance(first, int) else pl.multiple_of(start, TILE), count * TILE)


def _to_words(x):
    return pltpu.bitcast(x.astype(jnp.bfloat16), I32)


def _from_words(words):
    return pltpu.bitcast(words, jnp.bfloat16)


def _swap_bytes(a, b):
    x = (shr(a, _c(8)) ^ b) & _c(0x00FF00FF)
    return a ^ shl(x, _c(8)), b ^ x


def _choose_scale(w1, w2):
    magnitudes = sum((w & _c(0x7FFF)) + (shr(w, _c(16)) & _c(0x7FFF)) for w in (w1, w2))
    mean = jnp.sum(magnitudes.astype(jnp.float32)) * (0.25 / w1.size)
    return shr(mean.astype(I32) + _c(469), _c(1)) & _c(0x3FFF)


def _scale_terms(low, scale):
    d = (shr(low, _c(1)) & _bytes(0x7F)) + (_c(0x7F) - (scale & _c(0x7F))) * _bytes(0x01)
    base = (shr(scale, _c(7)) | _c(0x80)) * _bytes(0x01) - (shr(d, _c(7)) & _bytes(0x01))
    x = shr(d, _c(4)) & _bytes(0x07)
    return base, x + (shr(_bytes(0x08) - x, _c(3)) & _bytes(0x01)) + _bytes(0x80)


def _swap_zero_class(u, scale):
    zero = shr(scale, _c(7)) * _bytes(0x01)
    hit = (_bytes(0x80) - (u ^ zero)) | (_bytes(0x80) - (u ^ _bytes(ZERO)))
    hit = hit & _bytes(0x80)
    return u ^ ((hit - shr(hit, _c(7))) & (zero ^ _bytes(ZERO)))


def _to_ranks(low, high, scale):
    base, r = _scale_terms(low, scale)
    u = _swap_zero_class((base - (high & _bytes(0x7F))) & _bytes(0x7F), scale)
    top = (_bytes(0x80) - u) & _bytes(0x80)
    ranks = u - (shr(r - u, _c(7)) & _bytes(0x01)) + ((r + _bytes(0x01)) & (top - shr(top, _c(7))))
    return ranks, high & _bytes(0x80)


def _from_ranks(low, signed_ranks, scale):
    base, r = _scale_terms(low, scale)
    q = signed_ranks & _bytes(0x7F)
    at_most = r - q
    below = at_most - _bytes(0x01)
    top = (at_most ^ below) & _bytes(0x80)
    u = q + (shr(below, _c(7)) & _bytes(0x01)) - (q & (top - shr(top, _c(7))))
    return ((base - _swap_zero_class(u, scale)) & _bytes(0x7F)) | (signed_ranks & _bytes(0x80))


def _with_scales(fn, low, other, scales, i, c0):
    cut = min(max(DETOUR - c0, 0) * TILE, low.shape[1])
    left = jnp.where(i == 0, scales[1], scales[0])
    parts = [
        fn(low[:, lo:hi], other[:, lo:hi], scale)
        for lo, hi, scale in ((0, cut, left), (cut, low.shape[1], scales[0]))
        if lo < hi
    ]
    return jax.tree.map(lambda *columns: jnp.concatenate(columns, axis=1), *parts)


def _shift_back(words, bits):
    other = _c(32) - bits
    middle = [shr(words[k], bits) | shl(words[k - 1], other) for k in range(1, len(words))]
    return [shr(words[0], bits)] + middle + [shl(words[-1], other)]


def _shift_forward(words, bits):
    other = _c(32) - bits
    return [shl(words[k], bits) | shr(words[k + 1], other) for k in range(len(words) - 1)]


def _push_ranks(words, ranks):
    lengths = ranks + _bytes(0x01)
    la, lb = lengths & _c(0xFF), shr(lengths, _c(24))
    lc, ld = shr(lengths, _c(8)) & _c(0xFF), shr(lengths, _c(16)) & _c(0xFF)
    code = shl(jnp.ones_like(lb), lb) | _c(1)
    code = shl(code, lc) | _c(1)
    code = shl(code, ld) | _c(1)
    bits = (la + lb) + (lc + ld)
    room = _c(32) - bits
    out = _shift_back(words, bits)[: len(words)]
    return [shl(code, room) | out[0]] + out[1:], bits, room


def _pop_ranks(words):
    x = words[0]
    qa = lax.clz(x)
    x = shl(shl(x, _c(1)), qa)
    qb = lax.clz(x)
    x = shl(shl(x, _c(1)), qb)
    qc = lax.clz(x)
    x = shl(shl(x, _c(1)), qc)
    qd = lax.clz(x)
    bits = (qa + qb) + (qc + _c(4)) + qd
    out = _shift_forward(words, bits) + [shl(words[-1], bits)]
    return out, (qa | shl(qb, _c(24))) | (shl(qc, _c(8)) | shl(qd, _c(16)))


def _bits_through(word, ones):
    skip = jnp.zeros_like(word) + _c(32)
    for step in (16, 8, 4, 2, 1):
        less = skip - _c(step)
        skip = jnp.where(lax.population_count(shr(word, less)) < ones, less, skip)
    return _c(33) - skip


def _merge_halves(words, bits, count, out_words):
    half = bits.shape[1] // 2
    front = bits[:, half:]
    moved = _shift_back([w[:, :half] for w in words], front & _c(31))
    least, most = count // 32, len(words)
    hit = {j: shr(front, _c(5)) == j for j in range(least + 1, most + 1)}
    zero = jnp.zeros_like(front)
    out = []
    for k in range(out_words):
        v = moved[k - least] if 0 <= k - least < len(moved) else zero
        for j in range(least + 1, most + 1):
            if 0 <= k - j < len(moved):
                v = jnp.where(hit[j], moved[k - j], v)
            elif v is not zero:
                v = jnp.where(hit[j], zero, v)
        out.append(v | words[k][:, half:] if k < len(words) else v)
    return out, bits[:, :half] + front


def _split_halves(words, count, out_words):
    first, last = (count - 1) // 32, out_words - 1
    zero = jnp.zeros_like(words[0])

    def word(k):
        return words[k] if k < len(words) else zero

    seen = zero
    for k in range(first):
        seen = seen + lax.population_count(words[k])
    wanted = count - seen
    window = [word(first + k) for k in range(out_words + 1)]
    for j in range(first + 1, last + 1):
        seen = seen + lax.population_count(words[j - 1])
        later = seen < count
        wanted = jnp.where(later, count - seen, wanted)
        window = [jnp.where(later, word(j + k), v) for k, v in enumerate(window)]
    second = _shift_forward(window, _bits_through(window[0], wanted))
    return [jnp.concatenate([second[k], words[k]], axis=1) for k in range(out_words)]


def _slot_index():
    return lax.broadcasted_iota(I32, (8, TILE), 0), lax.broadcasted_iota(I32, (8, TILE), 1)


def _from_previous(x, row):
    y = pltpu.roll(x, 1, 0)
    return jnp.where(row == 0, pltpu.roll(y, 1, 1), y)


def _from_next(x, row):
    y = pltpu.roll(x, 7, 0)
    return jnp.where(row == 7, pltpu.roll(y, TILE - 1, 1), y)


def _last_row(x):
    return jnp.broadcast_to(x[7:8, :], x.shape)


def _bits_taken(over, row):
    def join(early, late):
        return early[0] + late[0], jnp.maximum(late[1], early[1] + late[0])

    run = over, jnp.maximum(over, 0)
    for k in (1, 2, 4):
        both = join([pltpu.roll(v, k, 0) for v in run], run)
        run = [jnp.where(row >= k, a, b) for a, b in zip(both, run)]
    lanes = [_last_row(v) for v in run]
    for unit in (1, 8):
        window = lanes
        for k in range(1, 8):
            lanes = join([pltpu.roll(v, k * unit, 1) for v in window], lanes)
    before = pltpu.roll(lanes[1], 1, 1)
    after = jnp.maximum(run[1], before + run[0])
    return jnp.where(row == 0, before, pltpu.roll(after, 1, 0))


def _sum_of_earlier(x, row, lane):
    run = x
    for k in (1, 2, 4):
        run = run + jnp.where(row >= k, pltpu.roll(run, k, 0), 0)
    lanes = total = _last_row(run)
    for unit, count in ((1, 8), (8, 16)):
        window = lanes
        for k in range(1, count):
            lanes = lanes + jnp.where(lane >= k * unit, pltpu.roll(window, k * unit, 1), 0)
    return (lanes - total) + (run - x)


def _code_step(i, w1, w2, scales, msg, state, c0=0, nc=8):
    low, high = _swap_bytes(w1, w2)
    msg[:, _tiles(LOW + 8 * i + c0, nc)] = low
    ranks, signs = _with_scales(_to_ranks, low, high, scales(), i, c0)
    msg[:, _tiles(RANKS + 8 * i + c0, nc)] = ranks | signs
    cols = _tiles(c0, nc)
    words, bits, room = _push_ranks([state[k, :, cols] for k in range(3)], ranks)
    for k in range(3):
        state[k, :, cols] = words[k]
    state[3, :, cols] = shr(state[3, :, cols], _c(1)) | signs
    state[4, :, cols] = state[4, :, cols] + bits
    state[5, :, cols] = state[5, :, cols] | room


def _code_finish(scales, msg, state):
    words, signs, bits = [state[0], state[1], state[2]], state[3], state[4]
    misfit = state[5]
    for count, out_words in ((32, 5), (64, 9), (128, LONGEST)):
        misfit = misfit | (_c(32 * len(words)) - bits)
        half = misfit.shape[1] // 2
        misfit = misfit[:, :half] | misfit[:, half:]
        words, bits = _merge_halves(words, bits, count, out_words)
    row, lane = _slot_index()
    first = (row | lane) == 0
    head = jnp.where(first, _c(32), 0)
    over = bits + head - _c(32 * SLOT)
    taken = _bits_taken(over, row)
    again = _from_previous(jnp.maximum(taken + over, 0), row)
    start = head + taken
    misfit = misfit | (_c(32 * LONGEST) - bits) | (taken - again) | (_c(32 * SLOT - 1) - start)
    fits = jnp.max(shr(misfit, _c(31)).astype(jnp.float32)) == 0.0

    zero = jnp.zeros_like(bits)
    words = _shift_back(words, start & _c(31))
    for j in (1, 2, 4, 8):
        move = (start & _c(32 * j)) != 0
        here = words + [zero] * j
        there = [zero] * j + words
        words = [jnp.where(move, b, a) for a, b in zip(here[: 2 * SLOT], there)]
    spill = [_from_previous(w, row) for w in words[SLOT:]]
    ones = sum(lax.population_count(w) for w in spill)
    words = [a | b for a, b in zip(words[:SLOT], _shift_back(spill, head))]
    header = scales[0] | jnp.where(fits, _c(0), _c(1 << 14)) | shl(scales[1] - scales[0], _c(24))
    words[0] = jnp.where(first, header | shl(ones, _c(15)), words[0])
    msg[:, _tiles(WORDS, SLOT)] = jnp.concatenate(words, axis=1)
    msg[:, _tiles(SIGNS, 8)] = signs
    return fits


def _read_header(msg):
    word = msg[:, _tiles(WORDS, 1)][0, 0]
    scale = word & _c(0x3FFF)
    scales = scale, scale + lax.shift_right_arithmetic(word, _c(24))
    return scales, (word & _c(1 << 14)) == 0, shr(word, _c(15)) & _c(0x1FF)


def _expand_ranks(msg, ones_in_first):
    signs = msg[:, _tiles(SIGNS, 8)]
    row, lane = _slot_index()
    first = (row | lane) == 0
    head = jnp.where(first, _c(32), 0)
    words = [msg[:, _tiles(WORDS + k, 1)] for k in range(SLOT)]
    words[0] = jnp.where(first, _c(0), words[0])
    zero = jnp.zeros_like(head)
    seen = [zero]
    for w in words:
        seen.append(seen[-1] + lax.population_count(w))
    foreign = ones_in_first + _sum_of_earlier(UNIT - seen[-1], row, lane)
    words += [_from_next(w, row) for w in _shift_forward(words + [zero], head)]
    index, wanted = zero, foreign
    for k in range(1, SLOT):
        later = seen[k] < foreign
        index = jnp.where(later, k, index)
        wanted = jnp.where(later, foreign - seen[k], wanted)
    for j in (8, 4, 2, 1):
        move = (index & _c(j)) != 0
        words = [
            jnp.where(move, words[min(k + j, len(words) - 1)], words[k]) for k in range(LONGEST + j)
        ]
    words = _shift_forward(words, jnp.where(foreign == 0, head, _bits_through(words[0], wanted)))
    for count, out_words in ((128, 9), (64, 5), (32, 3)):
        words = _split_halves(words, count, out_words)

    def step(j, words):
        words, ranks = _pop_ranks(list(words))
        msg[:, _tiles(RANKS + 8 * (STEPS - 1 - j), 8)] = ranks | (shl(signs, j) & _bytes(0x80))
        return tuple(words)

    lax.fori_loop(0, STEPS, step, tuple(words))


def _decode_step(i, scales, msg, c0=0, nc=8):
    low, ranks = msg[:, _tiles(LOW + 8 * i + c0, nc)], msg[:, _tiles(RANKS + 8 * i + c0, nc)]
    return _swap_bytes(low, _with_scales(_from_ranks, low, ranks, scales, i, c0))


def _body(x_hbm, out, xv, tx, rx, state, side, load_sems, send_sems, recv_sems, side_sems, ready):
    me = lax.axis_index("i")
    own = me ^ shr(me, 1)

    def first(h):
        return me ^ (3 - 2 * h)

    def second(h):
        return me ^ (1 + 2 * h)

    def row0(h, unit):
        return (4 * h + (own ^ (3, 2 - h, 1 + h, 0)[unit])) * UNIT

    def slab_start(i):
        return i * SLAB if isinstance(i, int) else pl.multiple_of(i * SLAB, SLAB)

    def load(h, unit):
        rows = pl.ds(pl.multiple_of(row0(h, unit), UNIT), UNIT)
        return pltpu.make_async_copy(x_hbm.at[rows], xv.at[h, unit], load_sems.at[2 * unit + h])

    between = me & 1
    lead = jnp.where(me == 1, 1, 0)

    def load_slab(j, i, c0=0, nc=8):
        h, cols = lead ^ j, _tiles(c0, nc)
        rows = pl.ds(pl.multiple_of(row0(h, D) + slab_start(i), SLAB), SLAB)
        sem = load_sems.at[8 + 2 * i + j if c0 == 0 else 8 + 2 * STEPS]
        return pltpu.make_async_copy(
            x_hbm.at[rows, cols], xv.at[h, D, pl.ds(slab_start(i), SLAB), cols], sem
        )

    def signal_neighbours(sem):
        for h in range(2):
            pl.semaphore_signal(
                sem, inc=1, device_id=(first(h),), device_id_type=pl.DeviceIdType.MESH
            )

    opening = [
        (0, 0, DETOUR, 8 - DETOUR),
        (0, 0, 0, DETOUR),
        (1 - between, between, 0, 8),
        (between, 1 - between, 0, 8),
    ]
    load_slab(*opening[0]).start()
    barrier = pltpu.get_barrier_semaphore()
    pl.when(me != 2)(lambda: signal_neighbours(barrier))
    load_slab(*opening[1]).start()
    load_slab(*opening[2]).start()

    @pl.when(me == 2)
    def _():
        pl.semaphore_wait(barrier, 2)
        signal_neighbours(ready)

    def copy(h, msg, part, tile, tiles):
        if msg == END_D:
            src, device = rx.at[h, END_S], first(h)
        else:
            src = tx.at[h, (D, F, S, O, O)[msg]]
            device = (first, first, second, second, first)[msg](h)
        k = (h * 6 + msg) * PARTS + part
        cols = _tiles(tile, tiles)
        return pltpu.make_async_remote_copy(
            src.at[:, cols],
            rx.at[h, msg, :, cols],
            send_sems.at[k],
            recv_sems.at[k],
            device_id=(device,),
            device_id_type=pl.DeviceIdType.MESH,
        )

    def low_slab(h, msg, i):
        return copy(h, msg, jnp.where(i < SLABS_A[msg], LOW_A, LOW_B), LOW + 8 * i, 8)

    def low_part(h, msg, part):
        lo, hi = ((0, SLABS_A[msg]), (SLABS_A[msg], STEPS))[part]
        return copy(h, msg, part, LOW + 8 * lo, 8 * (hi - lo))

    def first_low_part(h, short, act):
        pl.when(short)(lambda: act(copy(h, IN_S, LOW_A, LOW + DETOUR, 8 * SLABS_A[IN_S] - DETOUR)))
        pl.when(jnp.logical_not(short))(lambda: act(low_part(h, IN_S, LOW_A)))

    def tail_pieces(h):
        return [copy(h, END_D, TAIL + k, LOW + a, n) for k, (a, n) in enumerate(TAIL_PIECES)]

    def head(h, msg):
        return copy(h, msg, HEAD, WORDS, 1)

    def rest(h, msg, fits, act):
        pl.when(fits)(lambda: act(copy(h, msg, REST, WORDS + 1, RANKS - WORDS - 1)))
        pl.when(jnp.logical_not(fits))(lambda: act(copy(h, msg, REST, RANKS, END - RANKS)))

    def detour(h):
        return pltpu.make_async_remote_copy(
            side.at[2],
            side.at[h],
            side_sems.at[2],
            side_sems.at[h],
            device_id=(second(h),),
            device_id_type=pl.DeviceIdType.MESH,
        )

    def start(c):
        c.start()

    def wait_recv(c):
        c.wait_recv()

    def wait_send(c):
        c.wait_send()

    def note(plain, h, msg, fits):
        return plain | shl(jnp.where(fits, 0, 1), h * 6 + msg)

    def fitted(plain, h, msg):
        return (shr(plain, h * 6 + msg) & 1) == 0

    def receive_rest(h, msg, landed=None):
        scales, fits, ones = _read_header(rx.at[h, msg])
        rest(h, msg, fits, wait_recv)
        if landed is not None:
            landed(fits)
        pl.when(fits)(lambda: _expand_ranks(rx.at[h, msg], ones))
        return scales, fits

    def receive(h, msg):
        if msg == IN_S:
            first_low_part(h, me == 0, wait_recv)
        else:
            low_part(h, msg, LOW_A).wait_recv()
        low_part(h, msg, LOW_B).wait_recv()
        head(h, msg).wait_recv()
        return receive_rest(h, msg)[0]

    def slab(h, unit, i, c0=0, nc=8):
        r, cols = slab_start(i), _tiles(c0, nc)
        return xv[h, unit, pl.ds(r, 16), cols], xv[h, unit, pl.ds(r + 16, 16), cols]

    def code(words_of, h, unit, each):
        sample = words_of(0)
        scale = _choose_scale(*(w[:, DETOUR * TILE :] for w in sample))
        apart = _choose_scale(*(w[:, : DETOUR * TILE] for w in sample)) - scale
        scales = scale, scale + jnp.clip(apart, -128, 127)
        state[0] = jnp.zeros(state.shape[1:], I32)

        @pl.loop(0, STEPS)
        def _(i):
            _code_step(i, *words_of(i), lambda: scales, tx.at[h, unit], state.at[0])
            each(i)

        return _code_finish(scales, tx.at[h, unit], state.at[0])

    def plus(values, h, msg, scales, i):
        words = _decode_step(i, scales, rx.at[h, msg])
        if msg == IN_S:
            missing = jnp.where((me == 0) & (i == 0), DETOUR * TILE, 0)
            col = lax.broadcasted_iota(I32, words[0].shape, 1)
            words = [jnp.where(col < missing, 0, w) for w in words]
        return [v + _from_words(w).astype(jnp.float32) for v, w in zip(values, words)]

    def emit(h, unit, i, words, c0=0, nc=8):
        r, cols = pl.multiple_of(row0(h, unit) + i * SLAB, SLAB), _tiles(c0, nc)
        out[pl.ds(r, 16), cols] = _from_words(words[0])
        out[pl.ds(r + 16, 16), cols] = _from_words(words[1])

    def emit_slabs(h, unit, msg, scales, lo, hi):
        @pl.loop(lo, hi)
        def _(i):
            emit(h, unit, i, _decode_step(i, scales, rx.at[h, msg]))

    state[...] = jnp.zeros(state.shape, I32)
    pl.when(between == 1)(lambda: pl.semaphore_wait(barrier, 1))
    chosen = [None, None]

    def diagonal_scales(j):
        return (jnp.where(j == 1, chosen[1], chosen[0]),) * 2

    for n, (j, i, c0, nc) in enumerate(opening):
        h = lead ^ j
        load_slab(j, i, c0, nc).wait()
        words = [_to_words(v) for v in slab(h, D, i, c0, nc)]

        def send_then_scales(n=n, j=j, h=h, i=i, c0=c0, nc=nc, words=words):
            goes = me == 2 if n == 1 else (me == 2) | ((between == 1) & (j == 0))
            pl.when(goes)(lambda: copy(h, IN_S, LOW_A, LOW + 8 * i + c0, nc).start())
            if n == 0:
                load_slab(*opening[3]).start()
                for k in range(3, 2 * STEPS):
                    load_slab(k & 1, k // 2).start()
                chosen[0] = _choose_scale(*words)
            elif n == 1:
                side[2] = jnp.concatenate(words, axis=1)
            elif n == 2:
                chosen[1] = _choose_scale(*words)
            else:
                chosen[1] = jnp.where(j == 1, _choose_scale(*words), chosen[1])
            return (chosen[0],) * 2 if n < 2 else diagonal_scales(j)

        _code_step(i, *words, send_then_scales, tx.at[h, D], state.at[j], c0, nc)

    @pl.when(between == 1)
    def _():
        pl.semaphore_wait(ready, 1)
        copy(lead ^ 1, IN_S, LOW_A, LOW, 8).start()
        detour(lead).start()

    @pl.when(me == 0)
    def _():
        for h in range(2):
            rx[h, IN_S, :, _tiles(LOW, DETOUR)] = jnp.zeros((8, DETOUR * TILE), I32)
        pl.semaphore_wait(barrier, 2)
        copy(0, IN_S, LOW_A, LOW, 16).start()
        copy(1, IN_S, LOW_A, LOW, 8).start()

    for unit in (F, S, O):
        for h in range(2):
            load(h, unit).start()

    @pl.loop(3, 2 * STEPS)
    def _(n):
        j, i = n & 1, shr(n, 1)
        h = lead ^ j
        load_slab(j, i).wait()
        words = map(_to_words, slab(h, D, i))
        _code_step(i, *words, lambda: diagonal_scales(j), tx.at[h, D], state.at[j])
        low_slab(h, IN_S, i).start()

    def finish_diagonal(j, plain):
        h = lead ^ j
        fits = _code_finish(diagonal_scales(j), tx.at[h, D], state.at[j])
        head(h, IN_S).start()
        rest(h, IN_S, fits, start)
        return note(plain, h, IN_S, fits)

    plain = lax.fori_loop(0, 2, finish_diagonal, _c(0))

    def for_first(h, plain):
        load(h, F).wait()

        @pl.when(me == 2)
        def _():
            detour(h).wait_recv()
            for k in range(2):
                at = (h, F, pl.ds(16 * k, 16), _tiles(0, DETOUR))
                extra = _from_words(side[h, :, _tiles(k * DETOUR, DETOUR)])
                xv[at] = xv[at] + extra.astype(jnp.float32)

        def each(i):
            pl.when((h == 0) | (i < SLABS_A[IN_O]))(lambda: low_slab(h, IN_O, i).start())

        fits = code(lambda i: [_to_words(v) for v in slab(h, F, i)], h, F, each)

        @pl.when(h == 0)
        def _():
            head(h, IN_O).start()
            rest(h, IN_O, fits, start)

        return note(plain, h, IN_O, fits)

    plain = lax.fori_loop(0, 2, for_first, plain)

    def for_second(h, plain):
        load(h, S).wait()
        scales = receive(h, IN_S)
        fits = code(
            lambda i: [_to_words(v) for v in plus(slab(h, S, i), h, IN_S, scales, i)],
            h,
            S,
            lambda i: low_slab(h, PART_O, i).start(),
        )
        head(h, PART_O).start()
        rest(h, PART_O, fits, start)

        @pl.when(h == 0)
        def _():
            low_part(1, IN_O, LOW_B).start()
            head(1, IN_O).start()
            rest(1, IN_O, fitted(plain, 1, IN_O), start)

        return note(plain, h, PART_O, fits)

    plain = lax.fori_loop(0, 2, for_second, plain)

    def for_all(h, plain):
        load(h, O).wait()
        scales_in = receive(h, IN_O)
        scales_part = receive(h, PART_O)

        def total(i):
            values = plus(slab(h, O, i), h, IN_O, scales_in, i)
            words = [_to_words(v) for v in plus(values, h, PART_O, scales_part, i)]
            emit(h, O, i, words)
            return words

        def each(i):
            for msg in (END_S, END_F):
                low_slab(h, msg, i).start()

        fits = code(total, h, O, each)
        for msg in (END_S, END_F):
            head(h, msg).start()
            rest(h, msg, fits, start)
            plain = note(plain, h, msg, fits)
        return plain

    plain = lax.fori_loop(0, 2, for_all, plain)

    def from_neighbours(h, plain):
        low_part(h, END_S, LOW_A).wait_recv()
        low_part(h, END_D, LOW_A).start()
        low_part(h, END_S, LOW_B).wait_recv()
        head(h, END_S).wait_recv()
        head(h, END_D).start()

        def pass_on(fits):
            rest(h, END_D, fits, start)
            for piece in tail_pieces(h):
                piece.start()

        scales, fits = receive_rest(h, END_S, pass_on)
        emit_slabs(h, S, END_S, scales, 0, STEPS)
        emit_slabs(h, F, END_F, receive(h, END_F), 0, STEPS)
        return note(plain, h, END_D, fits)

    plain = lax.fori_loop(0, 2, from_neighbours, plain)

    def sent(h, msg, low_parts):
        for c in low_parts + [head(h, msg)]:
            c.wait_send()
        rest(h, msg, fitted(plain, h, msg), wait_send)

    @pl.loop(0, 2)
    def _(h):
        first_low_part(h, (between == 1) & (h == lead), wait_send)
        sent(h, IN_S, [low_part(h, IN_S, LOW_B)])
        for msg in range(IN_O, END_D):
            sent(h, msg, [low_part(h, msg, LOW_A), low_part(h, msg, LOW_B)])

    pl.when(between == 1)(lambda: detour(lead).wait_send())

    def diagonal_ranks(j, last_two):
        h = lead ^ j
        low_part(h, END_D, LOW_A).wait_recv()
        head(h, END_D).wait_recv()
        scales = receive_rest(h, END_D)[0]
        emit_slabs(h, D, END_D, scales, 0, SLABS_A[END_D])
        return last_two[1], scales

    scales_of = lax.fori_loop(0, 2, diagonal_ranks, ((_c(0), _c(0)),) * 2)
    for k, (tile, tiles) in enumerate(TAIL_PIECES):
        if k == len(TAIL_PIECES) - 2:
            for h in range(2):
                sent(h, END_D, [low_part(h, END_D, LOW_A)] + tail_pieces(h))
        for j in range(2):
            h = lead ^ j
            copy(h, END_D, TAIL + k, LOW + tile, tiles).wait_recv()
            if tiles > 8:
                emit_slabs(h, D, END_D, scales_of[j], tile // 8, (tile + tiles) // 8)
            else:
                words = _decode_step(tile // 8, scales_of[j], rx.at[h, END_D], tile % 8, tiles)
                emit(h, D, tile // 8, words, tile % 8, tiles)


def pallas_dist_rs_then_ag_i_m2048_n1024_kernel(x: jax.Array):
    return pl.pallas_call(
        _body,
        out_shape=jax.ShapeDtypeStruct((ROWS, N), jnp.bfloat16),
        in_specs=[pl.BlockSpec(memory_space=pl.ANY)],
        out_specs=pl.BlockSpec(memory_space=pltpu.VMEM),
        scratch_shapes=[
            pltpu.VMEM((2, 4, UNIT, N), jnp.float32),
            pltpu.VMEM((2, 4, 8, END * TILE), I32),
            pltpu.VMEM((2, 6, 8, END * TILE), I32),
            pltpu.VMEM((2, 6, 8, N), I32),
            pltpu.VMEM((3, 8, 2 * DETOUR * TILE), I32),
            pltpu.SemaphoreType.DMA((9 + 2 * STEPS,)),
            pltpu.SemaphoreType.DMA((12 * PARTS,)),
            pltpu.SemaphoreType.DMA((12 * PARTS,)),
            pltpu.SemaphoreType.DMA((3,)),
            pltpu.SemaphoreType.REGULAR,
        ],
        compiler_params=pltpu.CompilerParams(
            collective_id=0,
            vmem_limit_bytes=64 * 2**20,
            disable_bounds_checks=True,
            disable_semaphore_checks=True,
        ),
    )(x)
```
